```python
import numpy as np

kernel_name = "dist_ag_xy_y_m65536_n1024"

def setup_inputs():
    return {"x": np.random.randn(131072, 1024).astype(np.float32)}

def reference(x: np.ndarray) -> np.ndarray:
    return x
```

```python
import functools
import jax
import jax.numpy as jnp
from jax import lax
from jax.experimental import pallas as pl
from jax.experimental.pallas import tpu as pltpu

MESH = pl.DeviceIdType.MESH

def make(R=256, NI=4, NS=4, NY=8, NX=8, NO=4, LAG_Y=2, LAG_X=2, own_direct=True, out_dtype=jnp.float32):
    def fn(x):
        M, N = x.shape
        H = M // 2
        C = H // R

        def body(x_ref, o_ref, in_buf, s_buf, y_buf, x_buf, oy_buf, ox_buf,
                 in_sem, own_sem, own2_sem, ysend, yrecv, xsend, xrecv, oy_sem, ox_sem, ycred, xcred):
            mx = lax.axis_index("x")
            my = lax.axis_index("y")
            ynb = (mx, 1 - my)
            xnb = (1 - mx, my)
            mine = mx * H
            other = (1 - mx) * H
            own0 = my * M
            rem0 = (1 - my) * M

            def rows(base, c):
                return pl.ds(pl.multiple_of(base + c * R, R), R)

            def load(c):
                return pltpu.make_async_copy(x_ref.at[rows(mine, c)], in_buf.at[c % NI], in_sem.at[c % NI])
            def store_own(c):
                return pltpu.make_async_copy(in_buf.at[c % NI], o_ref.at[rows(own0 + mine, c)], own_sem.at[c % NI])
            def own2(c):
                return pltpu.make_async_copy(x_ref.at[rows(other, c)], o_ref.at[rows(own0 + other, c)], own2_sem.at[c % NI])
            def ycopy(c):
                return pltpu.make_async_remote_copy(s_buf.at[c % NS], y_buf.at[c % NY], ysend.at[c % NS], yrecv.at[c % NY], device_id=ynb, device_id_type=MESH)
            def xcopy(c):
                return pltpu.make_async_remote_copy(y_buf.at[c % NY], x_buf.at[c % NX], xsend.at[c % NY], xrecv.at[c % NX], device_id=xnb, device_id_type=MESH)
            def store_y(c):
                return pltpu.make_async_copy(oy_buf.at[c % NO], o_ref.at[rows(rem0 + mine, c)], oy_sem.at[c % NO])
            def store_x(c):
                return pltpu.make_async_copy(ox_buf.at[c % NO], o_ref.at[rows(rem0 + other, c)], ox_sem.at[c % NO])

            for c in range(NI - 1):
                load(c).start()

            bar = pltpu.get_barrier_semaphore()
            for nb in (ynb, xnb):
                pl.semaphore_signal(bar, 1, device_id=nb, device_id_type=MESH)
            pl.semaphore_wait(bar, 2)

            def step(t, _):
                c = t
                @pl.when(c < C)
                def _():
                    load(c).wait()
                    store_own(c).start()
                    @pl.when(c >= NS)
                    def _():
                        ycopy(c - NS).wait_send()
                    s_buf[c % NS] = in_buf[c % NI].astype(jnp.bfloat16)
                    @pl.when(c >= NY)
                    def _():
                        pl.semaphore_wait(ycred.at[c % NY], 1)
                    ycopy(c).start()
                    @pl.when(c >= NI)
                    def _():
                        own2(c - NI).wait()
                    own2(c).start()
                    @pl.when(c + NI - 1 < C)
                    def _():
                        @pl.when(c >= 1)
                        def _():
                            store_own(c - 1).wait()
                        load(c + NI - 1).start()
                c = t - LAG_Y
                @pl.when((c >= 0) & (c < C))
                def _():
                    ycopy(c).wait_recv()
                    @pl.when(c >= NX)
                    def _():
                        pl.semaphore_wait(xcred.at[c % NX], 1)
                    xcopy(c).start()
                    @pl.when(c >= NO)
                    def _():
                        store_y(c - NO).wait()
                    oy_buf[c % NO] = y_buf[c % NY].astype(jnp.float32)
                    store_y(c).start()
                c = t - LAG_Y - LAG_X
                @pl.when((c >= 0) & (c < C))
                def _():
                    xcopy(c).wait_send()
                    @pl.when(c + NY < C)
                    def _():
                        pl.semaphore_signal(ycred.at[c % NY], 1, device_id=ynb, device_id_type=MESH)
                    xcopy(c).wait_recv()
                    @pl.when(c >= NO)
                    def _():
                        store_x(c - NO).wait()
                    ox_buf[c % NO] = x_buf[c % NX].astype(jnp.float32)
                    store_x(c).start()
                    @pl.when(c + NX < C)
                    def _():
                        pl.semaphore_signal(xcred.at[c % NX], 1, device_id=xnb, device_id_type=MESH)
            lax.fori_loop(0, C + LAG_Y + LAG_X, step, None)

            for c in range(C - NI, C):
                store_own(c).wait()
                own2(c).wait()
            for c in range(C - NS, C):
                ycopy(c).wait_send()
            for c in range(C - NO, C):
                store_y(c).wait()
                store_x(c).wait()

        DMA = pltpu.SemaphoreType.DMA
        REG = pltpu.SemaphoreType.REGULAR
        return pl.pallas_call(
            body,
            out_shape=jax.ShapeDtypeStruct((2 * M, N), x.dtype),
            in_specs=[pl.BlockSpec(memory_space=pl.ANY)],
            out_specs=pl.BlockSpec(memory_space=pl.ANY),
            scratch_shapes=[
                pltpu.VMEM((NI, R, N), jnp.float32),
                pltpu.VMEM((NS, R, N), jnp.bfloat16),
                pltpu.VMEM((NY, R, N), jnp.bfloat16),
                pltpu.VMEM((NX, R, N), jnp.bfloat16),
                pltpu.VMEM((NO, R, N), jnp.float32),
                pltpu.VMEM((NO, R, N), jnp.float32),
                DMA((NI,)), DMA((NI,)), DMA((NI,)),
                DMA((NS,)), DMA((NY,)), DMA((NY,)), DMA((NX,)),
                DMA((NO,)), DMA((NO,)), REG((NY,)), REG((NX,)),
            ],
            compiler_params=pltpu.CompilerParams(collective_id=0, vmem_limit_bytes=100 * 1024 * 1024),
        )(x)
    return fn


def pallas_dist_ag_xy_y_m65536_n1024_kernel(x):
    return make()(x)
```

```python
import jax
import jax.numpy as jnp
import numpy as np
from jax import lax
from jax.experimental import pallas as pl
from jax.experimental.pallas import tpu as pltpu

def _i32(v):
    return np.int32(np.uint32(v).view(np.int32))

shl = lax.shift_left
shr = lax.shift_right_logical

SIGNS = _i32(0x80008000)
MAGS = _i32(0x7FFF7FFF)
EVEN = _i32(0x00FF00FF)
ODD = _i32(0xFF00FF00)
ONES = _i32(0x01010101)
TOP = _i32(0x80000000)

def c(x, v):
    return jnp.full(x.shape, v, jnp.int32)

def byte_sum(z):
    s = z + shr(z, c(z, 16))
    s = s + shr(s, c(s, 8))
    return s & 0xFF

def encode(words, top, buf, fill):
    lows, quads = [], []
    seen = None
    for a, b in zip(words[0::2], words[1::2]):
        ta = top - (a & MAGS)
        tb = top - (b & MAGS)
        lows.append((ta & EVEN) | (shl(tb, c(tb, 8)) & ODD))
        j = (shr(ta, c(ta, 8)) & EVEN) | (tb & ODD)
        seen = j if seen is None else seen | j
        ge4 = shr(j + _i32(0x7C7C7C7C), c(j, 7)) & ONES
        eq0 = shr(_i32(0x80808080) - j, c(j, 5)) & _i32(0x04040404)
        quads.append(j + ge4 + eq0 - ONES)
    signs = words[0] & SIGNS
    for k in range(1, 16):
        signs = signs | shr(words[k] & SIGNS, c(signs, k))
    stream = []
    longest = None
    for g in range(2):
        hi = lo = None
        total = fill
        for q in reversed(range(4)):
            z = quads[4 * g + q]
            n = byte_sum(z) + 4
            longest = n if longest is None else jnp.maximum(longest, n)
            total = total + n
            if hi is not None:
                n = n & 31
                spill = shl(hi, (32 - n) & 31)
                lo = spill if lo is None else shr(lo, n) | spill
            for k in reversed(range(4)):
                zk = (shr(z, c(z, 8 * k)) if k else z) & 31
                hi = c(z, TOP) if hi is None else shr(hi, c(hi, 1)) | TOP
                hi = shr(hi, zk)
        stream.append(buf | shr(hi, fill))
        buf = shr(lo, fill) | shl(shl(hi, c(hi, 1)), fill ^ 31)
        fill = jnp.maximum(total - 32, 0)
        longest = jnp.maximum(longest, fill)
        fill = fill & 31
    bad = (seen & _i32(0xE0E0E0E0)) | (longest & _i32(0xFFFFFFE0))
    return lows, signs, stream, buf, fill, bad

def decode(lows, signs, stream, top, fill):
    quads = []
    for g in range(2):
        w0, w1 = stream[g], stream[g + 1]
        hi = shl(w0, fill) | shr(shr(w1, c(w1, 1)), fill ^ 31)
        lo = shl(w1, fill)
        total = fill
        for q in range(4):
            z = n = None
            for k in range(4):
                zk = lax.clz(hi)
                step = zk + 1
                n = step if n is None else n + step
                z = zk if z is None else z | shl(zk, c(zk, 8 * k))
                if not (q == 3 and k == 3):
                    hi = shl(hi, step)
            quads.append(z)
            total = total + n
            if q < 3:
                hi = hi | shr(lo, 32 - n)
            if q < 2:
                lo = shl(lo, n)
        fill = jnp.maximum(total - 32, 0)
    words = []
    for i in range(8):
        z = quads[i]
        ge3 = (z + _i32(0x7D7D7D7D)) & _i32(0x80808080)
        ge4 = (z + _i32(0x7C7C7C7C)) & _i32(0x80808080)
        j = z + ONES + shr(ge4, c(z, 5)) - shr(ge4, c(z, 7)) - shr(ge3, c(z, 5))
        ta = (lows[i] & EVEN) | (shl(j, c(j, 8)) & ODD)
        tb = (shr(lows[i], c(j, 8)) & EVEN) | (j & ODD)
        for k, t in ((2 * i, ta), (2 * i + 1, tb)):
            s = (shl(signs, c(t, k)) if k else signs) & SIGNS
            words.append((top - t) | s)
    return words, fill


MESH = pl.DeviceIdType.MESH
R = 256
MAIN, SLOT = 11, 18

def make(NI=3, NS=2, NY=4, NX=4, HB=36, BR=512):
    def fn(x):
        M, N = x.shape
        H = M // 2
        C = H // R
        PER = BR // R
        NB = H // BR
        VB = NB - HB
        CH = HB * PER

        def body(x_ref, oh_ref, ov_ref, in_buf, s_buf, y_buf, x_buf, state, raw,
                 in_sem, out_sem, ysend, yrecv, xsend, xrecv, ycred, xcred):
            mx = lax.axis_index("x")
            my = lax.axis_index("y")
            ynb = (mx, 1 - my)
            xnb = (1 - mx, my)
            halves = (mx, 1 - mx)
            quarter = (2 * my + mx, 2 * my + 1 - mx, 2 * (1 - my) + mx, 2 * (1 - my) + 1 - mx)

            def load(h, c):
                rows = pl.ds(pl.multiple_of(halves[h] * H + c * R, R), R)
                return pltpu.make_async_copy(x_ref.at[rows], in_buf.at[h, c % NI], in_sem.at[h, c % NI])

            def rows_of(c):
                return pl.ds(pl.multiple_of((c % PER) * R, R), R)

            def result(s, c):
                blk = jnp.where(c < CH, VB - 1, (c - CH) // PER)
                return ov_ref.at[quarter[s], blk, rows_of(c)]

            def spill(s, c):
                return pltpu.make_async_copy(ov_ref.at[quarter[s], VB - 1, rows_of(c)],
                                             oh_ref.at[quarter[s], c // PER, rows_of(c)], out_sem.at[s, c % PER])

            def before_result(s, c):
                @pl.when((c >= PER) & (c < CH + PER))
                def _():
                    spill(s, c - PER).wait()

            def after_result(s, c):
                @pl.when(c < CH)
                def _():
                    spill(s, c).start()

            PARTS = (pl.ds(0, MAIN), pl.ds(MAIN, SLOT - MAIN), pl.ds(0, 1))
            def ycopy(c, part):
                k = part % 2
                return pltpu.make_async_remote_copy(s_buf.at[c % NS, PARTS[part]], y_buf.at[c % NY, PARTS[part]],
                                                    ysend.at[k, c % NS], yrecv.at[k, c % NY], device_id=ynb, device_id_type=MESH)
            def xcopy(c, part):
                k = part % 2
                return pltpu.make_async_remote_copy(y_buf.at[c % NY, PARTS[part]], x_buf.at[c % NX, PARTS[part]],
                                                    xsend.at[k, c % NY], xrecv.at[k, c % NX], device_id=xnb, device_id_type=MESH)

            def top_word(e):
                half = shl(e, jnp.full_like(e, 7)) | 0x7F
                return half | shl(half, jnp.full_like(e, 16))

            def is_raw(buf, slot):
                return jnp.max(jnp.where(buf[slot, 1, :, 0:128] == 0, 1, 0))

            def unpack(s, buf, n, c, st):
                slot = c % n
                dst = result(s, c)
                @pl.when(c == 0)
                def _():
                    w = buf[0, 0]
                    state[st] = jnp.full_like(w, 8)
                    state[st + 1] = top_word(shr(w, jnp.full_like(w, 24)))
                before_result(s, c)
                flag = raw[s - 1, slot]
                @pl.when(flag == 0)
                def _():
                    words, fill = decode([buf[slot, 3 + i] for i in range(8)], buf[slot, 2],
                                               [buf[slot, 0], buf[slot, 1], buf[(c + 1) % n, 0]], state[st + 1], state[st])
                    state[st] = fill
                    for k in range(16):
                        dst[pl.ds(16 * k, 16), :] = pltpu.bitcast(words[k], jnp.bfloat16)
                @pl.when(flag != 0)
                def _():
                    state[st] = jnp.zeros((8, N), jnp.int32)
                    for k in range(16):
                        dst[pl.ds(16 * k, 16), :] = pltpu.bitcast(buf[slot, 2 + k], jnp.bfloat16)
                after_result(s, c)

            for c in range(NI):
                load(0, c).start()
                load(1, c).start()

            bar = pltpu.get_barrier_semaphore()
            for nb in (ynb, xnb):
                pl.semaphore_signal(bar, 1, device_id=nb, device_id_type=MESH)
            pl.semaphore_wait(bar, 2)

            def step(t, _):
                c = t
                @pl.when((c >= NS) & (c < C + NS))
                def _():
                    ycopy(c - NS, 0).wait_send()
                    @pl.when(raw[0, c % NS] != 0)
                    def _():
                        ycopy(c - NS, 1).wait_send()

                @pl.when(c < C)
                def _():
                    slot = c % NS
                    load(0, c).wait()
                    before_result(0, c)
                    dst = result(0, c)
                    src = in_buf.at[0, c % NI]
                    @pl.when(c == 0)
                    def _():
                        w = pltpu.bitcast(src[0:16, :].astype(jnp.bfloat16), jnp.int32)
                        e = (shr(w, jnp.full_like(w, 7)) & 0xFF) + (shr(w, jnp.full_like(w, 23)) & 0xFF)
                        top = jnp.minimum(jnp.sum(e) // (16 * N) + 4, 255)
                        top = jnp.full_like(w, top)
                        state[0] = shl(top, jnp.full_like(w, 24))
                        state[1] = jnp.full_like(w, 8)
                        state[2] = top_word(top)
                    words = []
                    for k in range(16):
                        b = src[pl.ds(16 * k, 16), :].astype(jnp.bfloat16)
                        dst[pl.ds(16 * k, 16), :] = b
                        words.append(pltpu.bitcast(b, jnp.int32))
                    lows, signs, stream, carry, fill, bad = encode(words, state[2], state[0], state[1])
                    for i, v in enumerate(stream + [signs] + lows):
                        s_buf[slot, i] = v
                    state[0] = carry
                    state[1] = fill
                    flag = jnp.max(jnp.where(bad != 0, 1, 0))
                    raw[0, slot] = flag
                    @pl.when(flag != 0)
                    def _():
                        zero = jnp.zeros((8, N), jnp.int32)
                        state[0] = zero
                        state[1] = zero
                        s_buf[slot, 1] = zero
                        for k in range(16):
                            s_buf[slot, 2 + k] = pltpu.bitcast(src[pl.ds(16 * k, 16), :].astype(jnp.bfloat16), jnp.int32)
                    @pl.when(c >= NY)
                    def _():
                        pl.semaphore_wait(ycred.at[c % NY], 1)
                    ycopy(c, 0).start()
                    @pl.when(flag != 0)
                    def _():
                        ycopy(c, 1).start()
                    after_result(0, c)

                    load(1, c).wait()
                    before_result(1, c)
                    result(1, c)[...] = in_buf[1, c % NI].astype(jnp.bfloat16)
                    after_result(1, c)
                    @pl.when(c + NI < C)
                    def _():
                        load(0, c + NI).start()
                        load(1, c + NI).start()

                @pl.when(c == C)
                def _():
                    s_buf[C % NS, 0] = state[0]
                    pl.semaphore_wait(ycred.at[C % NY], 1)
                    ycopy(C, 2).start()

                c = t - 1
                @pl.when((c >= 0) & (c < C))
                def _():
                    ycopy(c, 0).wait_recv()
                    @pl.when(c >= NX)
                    def _():
                        pl.semaphore_wait(xcred.at[c % NX], 1)
                    xcopy(c, 0).start()
                    flag = is_raw(y_buf, c % NY)
                    raw[1, c % NY] = flag
                    @pl.when(flag != 0)
                    def _():
                        ycopy(c, 1).wait_recv()
                        xcopy(c, 1).start()
                @pl.when(c == C)
                def _():
                    ycopy(C, 2).wait_recv()
                    pl.semaphore_wait(xcred.at[C % NX], 1)
                    xcopy(C, 2).start()

                c = t - 2
                @pl.when((c >= 0) & (c < C))
                def _():
                    unpack(2, y_buf, NY, c, 3)
                    xcopy(c, 0).wait_recv()
                    flag = is_raw(x_buf, c % NX)
                    raw[2, c % NX] = flag
                    @pl.when(flag != 0)
                    def _():
                        xcopy(c, 1).wait_recv()
                @pl.when(c == C)
                def _():
                    xcopy(C, 2).wait_recv()

                c = t - 3
                @pl.when(c >= 0)
                def _():
                    unpack(3, x_buf, NX, c, 5)
                    @pl.when(c + NX <= C)
                    def _():
                        pl.semaphore_signal(xcred.at[c % NX], 1, device_id=xnb, device_id_type=MESH)

                c = t - 2
                @pl.when((c >= 0) & (c < C))
                def _():
                    xcopy(c, 0).wait_send()
                    @pl.when(raw[1, c % NY] != 0)
                    def _():
                        xcopy(c, 1).wait_send()
                    @pl.when(c + NY <= C)
                    def _():
                        pl.semaphore_signal(ycred.at[c % NY], 1, device_id=ynb, device_id_type=MESH)
            lax.fori_loop(0, C + 3, step, None)
            ycopy(C, 2).wait_send()
            xcopy(C, 2).wait_send()

        DMA = pltpu.SemaphoreType.DMA
        REG = pltpu.SemaphoreType.REGULAR
        assert NS == 2
        oh, ov = pl.pallas_call(
            body,
            out_shape=[jax.ShapeDtypeStruct((4, HB, BR, N), jnp.bfloat16), pltpu.VMEM((4, VB, BR, N), jnp.bfloat16)],
            in_specs=[pl.BlockSpec(memory_space=pl.ANY)],
            out_specs=[pl.BlockSpec(memory_space=pl.ANY), pl.BlockSpec(memory_space=pltpu.VMEM)],
            scratch_shapes=[
                pltpu.VMEM((2, NI, R, N), jnp.float32),
                pltpu.VMEM((NS, SLOT, 8, N), jnp.int32),
                pltpu.VMEM((NY, SLOT, 8, N), jnp.int32),
                pltpu.VMEM((NX, SLOT, 8, N), jnp.int32),
                pltpu.VMEM((7, 8, N), jnp.int32),
                pltpu.SMEM((3, max(NS, NY, NX)), jnp.int32),
                DMA((2, NI)), DMA((4, PER)), DMA((2, NS)), DMA((2, NY)), DMA((2, NY)), DMA((2, NX)),
                REG((NY,)), REG((NX,)),
            ],
            compiler_params=pltpu.CompilerParams(collective_id=0),
        )(x)
        return jnp.concatenate([oh, ov], axis=1).reshape(2 * M, N)
    return fn


def pallas_dist_ag_xy_y_m65536_n1024_kernel(x):
    return make()(x)
```

```python
import contextlib
import jax
import jax.numpy as jnp
import numpy as np
from jax import lax
from jax.experimental import pallas as pl
from jax.experimental.pallas import tpu as pltpu

def _i32(v):
    return np.uint32(v).view(np.int32)

def shl(x, n):
    return lax.shift_left(x, jnp.full_like(x, n) if isinstance(n, int) else n)

def shr(x, n):
    return lax.shift_right_logical(x, jnp.full_like(x, n) if isinstance(n, int) else n)

SIGNS = _i32(0x80008000)
MAGS = _i32(0x7FFF7FFF)
EVEN = _i32(0x00FF00FF)
ODD = _i32(0xFF00FF00)
ONES = _i32(0x01010101)
TOP = _i32(0x80000000)

LANES = 256
GROUPS = 8
RATE = 28
WORDS = GROUPS * RATE // 32

def byte_sum(z):
    s = z + shr(z, 16)
    return (s + shr(s, 8)) & 0xFF

def block(x, b):
    return x[:, b * LANES:(b + 1) * LANES]

def encode(words, top, carry, fill):
    reach = len(carry)
    lows, quads = [], []
    seen = None
    for a, b in zip(words[0::2], words[1::2]):
        ta = top - (a & MAGS)
        tb = top - (b & MAGS)
        lows.append((ta & EVEN) | (shl(tb, 8) & ODD))
        j = (shr(ta, 8) & EVEN) | (tb & ODD)
        seen = j if seen is None else seen | j
        ge4 = shr(j + _i32(0x7C7C7C7C), 7) & ONES
        eq0 = shr(_i32(0x80808080) - j, 5) & _i32(0x04040404)
        quads.append(j + ge4 + eq0 - ONES)
    signs = words[0] & SIGNS
    for k in range(1, 16):
        signs = signs | shr(words[k] & SIGNS, k)
    strings = []
    longest = None
    for h in range(2):
        hi = lo = total = None
        for q in reversed(range(4)):
            z = quads[4 * h + q]
            n = byte_sum(z) + 4
            longest = n if longest is None else jnp.maximum(longest, n)
            total = n if total is None else total + n
            if hi is not None:
                n = n & 31
                spill = shl(hi, (32 - n) & 31)
                lo = spill if lo is None else shr(lo, n) | spill
            for k in reversed(range(4)):
                zk = (shr(z, 8 * k) if k else z) & 31
                hi = jnp.full_like(z, TOP) if hi is None else shr(hi, 1) | TOP
                hi = shr(hi, zk)
        longest = jnp.maximum(longest, shr(total, 1))
        strings.append((hi, lo, total))
    bad = (seen & _i32(0xE0E0E0E0)) | (longest & _i32(0xFFFFFFE0))

    out = list(carry) + [None] * WORDS
    pos = fill
    far = None
    for g in range(GROUPS):
        hi, lo, total = (block(v, g // 2) for v in strings[g % 2])
        first = RATE * g // 32
        start = jnp.maximum(pos, RATE * g) if g else pos
        pos = start + total
        skip = shr(start, 5) - first
        far = skip if far is None else jnp.maximum(far, skip)
        s = start & 31
        back = s ^ 31
        piece = [shr(hi, s), shl(shl(hi, 1), back) | shr(lo, s), shl(shl(lo, 1), back)]
        d = 1
        while d < reach:
            move = (skip & d) != 0
            width = min(len(piece) + d, reach + 2)
            piece = [jnp.where(move, piece[i - d] if i >= d else 0, piece[i] if i < len(piece) else 0) for i in range(width)]
            d *= 2
        for i, p in enumerate(piece):
            if first + i < len(out):
                out[first + i] = p if out[first + i] is None else out[first + i] | p
    fill = jnp.maximum(pos - 32 * WORDS, 0)
    far = jnp.maximum(far, shr(fill, 5))
    return lows, signs, out[:WORDS], out[WORDS:], fill, bad, far >= reach

def decode(lows, signs, stream, top, fill):
    reach = len(stream) - WORDS
    quads = [[None] * GROUPS for _ in range(4)]
    pos = fill
    for g in range(GROUPS):
        first = RATE * g // 32
        start = jnp.maximum(pos, RATE * g) if g else pos
        skip = shr(start, 5) - first
        piece = stream[first:first + reach + 2]
        d = 1 << (reach - 1).bit_length() - 1
        while d:
            move = (skip & d) != 0
            piece = [jnp.where(move, piece[i + d], piece[i]) if i + d < len(piece) else piece[i] for i in range(min(d + 2, len(piece)))]
            d //= 2
        s = start & 31
        back = s ^ 31
        hi = shl(piece[0], s) | shr(shr(piece[1], 1), back)
        lo = shl(piece[1], s) | shr(shr(piece[2], 1), back)
        pos = start
        for q in range(4):
            z = n = None
            for k in range(4):
                zk = lax.clz(hi)
                step = zk + 1
                n = step if n is None else n + step
                z = zk if z is None else z | shl(zk, 8 * k)
                if not (q == 3 and k == 3):
                    hi = shl(hi, step)
            quads[q][g] = z
            pos = pos + n
            if q < 3:
                hi = hi | shr(lo, 32 - n)
            if q < 2:
                lo = shl(lo, n)
    fill = jnp.maximum(pos - 32 * WORDS, 0)
    words = []
    for i in range(8):
        z = jnp.concatenate(quads[i % 4][i // 4::2], axis=1)
        ge3 = (z + _i32(0x7D7D7D7D)) & _i32(0x80808080)
        ge4 = (z + _i32(0x7C7C7C7C)) & _i32(0x80808080)
        j = z + ONES + shr(ge4, 5) - shr(ge4, 7) - shr(ge3, 5)
        ta = (lows[i] & EVEN) | (shl(j, 8) & ODD)
        tb = (shr(lows[i], 8) & EVEN) | (j & ODD)
        for k, t in ((2 * i, ta), (2 * i + 1, tb)):
            s = (shl(signs, k) if k else signs) & SIGNS
            words.append((top - t) | s)
    return words, fill


MESH = pl.DeviceIdType.MESH
R = 256

def make(NI=3, NS=2, NY=4, NX=4, REACH=5, CUTS=(11, 22, 33), first_alone=False, order=None, scopes=False, late_barrier=True, cp={}):
    MAIN = WORDS + 4 + 32
    SLOT = WORDS + 64
    edges = (0,) + tuple(CUTS) + (MAIN,)
    P = len(edges) - 1
    def fn(x):
        M, N = x.shape
        H = M // 2
        C = H // R
        G = R // 2
        SEG, FAR, NEAR = 2048, 9, 7
        SEGS = H // SEG
        CH = SEGS * FAR // 2
        PER = 2

        def body(x_ref, oh_ref, ov_ref, in_buf, s_buf, y_buf, x_buf, carry_ref, fill_ref, top_ref, raw,
                 in_sem, out_sem, ysend, yrecv, xsend, xrecv, ycred, xcred):
            mx = lax.axis_index("x")
            my = lax.axis_index("y")
            ynb = (mx, 1 - my)
            xnb = (1 - mx, my)
            halves = (mx, 1 - mx)
            quarter = (2 * my + mx, 2 * my + 1 - mx, 2 * (1 - my) + mx, 2 * (1 - my) + 1 - mx)

            def piece(i):
                return pl.ds(pl.multiple_of(i * G, G), G)

            def load_piece(h, c, i):
                u = 2 * c + i
                v = jnp.maximum(u - 2 * CH, 0)
                first = jnp.where(c < CH, (u // FAR) * (FAR + NEAR) + u % FAR, (v // NEAR) * (FAR + NEAR) + FAR + v % NEAR)
                return pltpu.make_async_copy(x_ref.at[piece(halves[h] * (H // G) + first)], in_buf.at[h, c % NI, piece(i)], in_sem.at[h, c % NI])

            class load:
                def __init__(self, h, c):
                    self.h, self.c = h, c
                def start(self):
                    for i in range(2):
                        load_piece(self.h, self.c, i).start()
                def wait(self):
                    whole = in_buf.at[self.h, self.c % NI]
                    pltpu.make_async_copy(whole, whole, in_sem.at[self.h, self.c % NI]).wait()

            def result(s, c, i):
                v = 2 * jnp.where(c < CH, C - PER + c % PER - CH, c - CH) + i
                return ov_ref.at[quarter[s] * SEGS + v // NEAR, piece(v % NEAR)]

            def spill(s, c, i):
                u = 2 * c + i
                return pltpu.make_async_copy(result(s, c, i), oh_ref.at[quarter[s] * SEGS + u // FAR, piece(u % FAR)], out_sem.at[s, c % PER, i])

            def before_result(s, c):
                @pl.when((c >= PER) & (c < CH + PER))
                def _():
                    for i in range(2):
                        spill(s, c - PER, i).wait()

            def after_result(s, c):
                @pl.when(c < CH)
                def _():
                    for i in range(2):
                        spill(s, c, i).start()

            def put(s, c, blocks):
                dst = [result(s, c, i) for i in range(2)]
                for k, b in enumerate(blocks):
                    dst[k // 8][pl.ds(16 * (k % 8), 16), :] = b

            def lanes(first, count=1):
                return pl.ds(first * LANES, count * LANES)

            PARTS = [lanes(a, b - a) for a, b in zip(edges, edges[1:])] + [lanes(MAIN, SLOT - MAIN), lanes(0, REACH)]
            def ycopy(c, part):
                k = part % (P + 1)
                return pltpu.make_async_remote_copy(s_buf.at[c % NS, :, PARTS[part]], y_buf.at[c % NY, :, PARTS[part]],
                                                    ysend.at[k, c % NS], yrecv.at[k, c % NY], device_id=ynb, device_id_type=MESH)
            def xcopy(c, part):
                k = part % (P + 1)
                return pltpu.make_async_remote_copy(y_buf.at[c % NY, :, PARTS[part]], x_buf.at[c % NX, :, PARTS[part]],
                                                    xsend.at[k, c % NY], xrecv.at[k, c % NX], device_id=xnb, device_id_type=MESH)

            def top_word(e):
                half = shl(e, 7) | 0x7F
                return half | shl(half, 16)

            def is_raw(buf, slot):
                return jnp.max(jnp.where(buf[slot, :, pl.ds((WORDS - 1) * LANES, 128)] == 0, 1, 0))

            def unpack(s, buf, n, c):
                slot = c % n
                @pl.when(c == 0)
                def _():
                    top = top_word(shr(buf[0, :, lanes(0)], 24))
                    fill_ref[s - 1] = jnp.full_like(top, 8)
                    top_ref[s - 1] = jnp.concatenate([top] * (N // LANES), axis=1)
                before_result(s, c)
                flag = raw[s - 1, slot]
                @pl.when(flag == 0)
                def _():
                    stream = [buf[slot, :, lanes(i)] for i in range(WORDS)] + [buf[(c + 1) % n, :, lanes(i)] for i in range(REACH)]
                    words, fill = decode([buf[slot, :, lanes(WORDS + 4 + 4 * i, 4)] for i in range(8)], buf[slot, :, lanes(WORDS, 4)],
                                               stream, top_ref[s - 1], fill_ref[s - 1])
                    fill_ref[s - 1] = fill
                    put(s, c, [pltpu.bitcast(w, jnp.bfloat16) for w in words])
                @pl.when(flag != 0)
                def _():
                    fill_ref[s - 1] = jnp.zeros((8, LANES), jnp.int32)
                    put(s, c, [pltpu.bitcast(buf[slot, :, lanes(WORDS + 4 * k, 4)], jnp.bfloat16) for k in range(16)])
                after_result(s, c)

            load(0, 0).start()
            if not first_alone:
                for c in range(1, NI):
                    load(0, c).start()
                    load(1, c - 1).start()
                load(1, NI - 1).start()

            bar = pltpu.get_barrier_semaphore()
            for nb in (ynb, xnb):
                pl.semaphore_signal(bar, 1, device_id=nb, device_id_type=MESH)
            if not late_barrier:
                pl.semaphore_wait(bar, 2)

            def pack(c):
                @pl.when((c >= NS) & (c < C + NS))
                def _():
                    for p in range(P):
                        ycopy(c - NS, p).wait_send()
                    @pl.when(raw[0, c % NS] != 0)
                    def _():
                        ycopy(c - NS, P).wait_send()

                @pl.when(c < C)
                def _():
                    slot = c % NS
                    load(0, c).wait()
                    before_result(0, c)
                    src = in_buf.at[0, c % NI]
                    @pl.when(c == 0)
                    def _():
                        if first_alone:
                            load(1, 0).start()
                            for i in range(1, NI):
                                load(0, i).start()
                                load(1, i).start()
                        w = pltpu.bitcast(src[0:16, :].astype(jnp.bfloat16), jnp.int32)
                        e = (shr(w, 7) & 0xFF) + (shr(w, 23) & 0xFF)
                        top = jnp.full_like(w, jnp.minimum(jnp.sum(e) // (16 * N) + 4, 255))
                        carry_ref[0] = shl(top[:, :LANES], 24)
                        for i in range(1, REACH):
                            carry_ref[i] = jnp.zeros((8, LANES), jnp.int32)
                        fill_ref[0] = jnp.full((8, LANES), 8, jnp.int32)
                        top_ref[0] = top_word(top)
                    rounded = [src[pl.ds(16 * k, 16), :].astype(jnp.bfloat16) for k in range(16)]
                    put(0, c, rounded)
                    words = [pltpu.bitcast(b, jnp.int32) for b in rounded]
                    carry = [carry_ref[i] for i in range(REACH)]
                    lows, signs, stream, ncarry, fill, bad, far = encode(words, top_ref[0], carry, fill_ref[0])
                    for i, v in enumerate(stream):
                        s_buf[slot, :, lanes(i)] = v
                    for i, v in enumerate([signs] + lows):
                        s_buf[slot, :, lanes(WORDS + 4 * i, 4)] = v
                    for i, v in enumerate(ncarry):
                        carry_ref[i] = v
                    fill_ref[0] = fill
                    flag = jnp.where(far, 1, 0)
                    for b in range(N // LANES):
                        flag = flag | block(bad, b)
                    flag = jnp.max(jnp.where(flag != 0, 1, 0))
                    raw[0, slot] = flag
                    @pl.when(flag != 0)
                    def _():
                        zero = jnp.zeros((8, LANES), jnp.int32)
                        fill_ref[0] = zero
                        for i in range(WORDS):
                            s_buf[slot, :, lanes(i)] = carry[i] if i < REACH else zero
                        for i in range(REACH):
                            carry_ref[i] = zero
                        for k in range(16):
                            s_buf[slot, :, lanes(WORDS + 4 * k, 4)] = pltpu.bitcast(src[pl.ds(16 * k, 16), :].astype(jnp.bfloat16), jnp.int32)
                    if late_barrier:
                        @pl.when(c == 0)
                        def _():
                            pl.semaphore_wait(bar, 2)
                    @pl.when(c >= NY)
                    def _():
                        pl.semaphore_wait(ycred.at[c % NY], 1)
                    for p in range(P):
                        ycopy(c, p).start()
                    @pl.when(flag != 0)
                    def _():
                        ycopy(c, P).start()
                    after_result(0, c)

                @pl.when(c == C)
                def _():
                    for i in range(REACH):
                        s_buf[C % NS, :, lanes(i)] = carry_ref[i]
                    pl.semaphore_wait(ycred.at[C % NY], 1)
                    ycopy(C, P + 1).start()

            def own(c):
                @pl.when(c < C)
                def _():
                    load(1, c).wait()
                    before_result(1, c)
                    for i in range(2):
                        result(1, c, i)[...] = in_buf[1, c % NI, piece(i)].astype(jnp.bfloat16)
                    after_result(1, c)
                    @pl.when(c + NI < C)
                    def _():
                        load(0, c + NI).start()
                        load(1, c + NI).start()

            def forward(c, p):
                @pl.when((c >= 0) & (c < C))
                def _():
                    ycopy(c, p).wait_recv()
                    if p == 0:
                        @pl.when(c >= NX)
                        def _():
                            pl.semaphore_wait(xcred.at[c % NX], 1)
                    xcopy(c, p).start()
                    if p == 0:
                        raw[1, c % NY] = is_raw(y_buf, c % NY)
                    if p == P - 1:
                        @pl.when(raw[1, c % NY] != 0)
                        def _():
                            ycopy(c, P).wait_recv()
                            xcopy(c, P).start()
                if p == 0:
                    @pl.when(c == C)
                    def _():
                        ycopy(C, P + 1).wait_recv()
                        pl.semaphore_wait(xcred.at[C % NX], 1)
                        xcopy(C, P + 1).start()

            def unpack_y(c):
                @pl.when((c >= 0) & (c < C))
                def _():
                    unpack(2, y_buf, NY, c)

            def release_y(c):
                @pl.when((c >= 0) & (c < C))
                def _():
                    for p in range(P):
                        xcopy(c, p).wait_send()
                    @pl.when(raw[1, c % NY] != 0)
                    def _():
                        xcopy(c, P).wait_send()
                    @pl.when(c + NY <= C)
                    def _():
                        pl.semaphore_signal(ycred.at[c % NY], 1, device_id=ynb, device_id_type=MESH)

            def unpack_x(c):
                @pl.when((c >= 0) & (c < C))
                def _():
                    for p in range(1, P):
                        xcopy(c, p).wait_recv()
                    @pl.when(raw[2, c % NX] != 0)
                    def _():
                        xcopy(c, P).wait_recv()
                @pl.when((c >= -1) & (c < C - 1))
                def _():
                    xcopy(c + 1, 0).wait_recv()
                    raw[2, (c + 1) % NX] = is_raw(x_buf, (c + 1) % NX)
                @pl.when(c == C - 1)
                def _():
                    xcopy(C, P + 1).wait_recv()
                @pl.when((c >= 0) & (c < C))
                def _():
                    unpack(3, x_buf, NX, c)
                    @pl.when(c + NX <= C)
                    def _():
                        pl.semaphore_signal(xcred.at[c % NX], 1, device_id=xnb, device_id_type=MESH)

            seq = order or {1: "p f y o x r", 2: "p f y o f x r", 3: "p f y o f x f r", 4: "p f y f x f o r f"}[P]
            def step(t, _):
                part = 0
                for s in seq.split():
                  with (jax.named_scope(s + str(part)) if scopes else contextlib.nullcontext()):
                    if s == "p": pack(t)
                    elif s == "o": own(t)
                    elif s == "f":
                        forward(t - 1, part); part += 1
                    elif s == "y": unpack_y(t - 2)
                    elif s == "x": unpack_x(t - 2)
                    elif s == "X": unpack_x(t - 3)
                    elif s == "r": release_y(t - 2)
                assert part == P
            lax.fori_loop(0, C + (3 if "X" in seq else 2), step, None)
            ycopy(C, P + 1).wait_send()
            xcopy(C, P + 1).wait_send()

        DMA = pltpu.SemaphoreType.DMA
        REG = pltpu.SemaphoreType.REGULAR
        assert NS == 2
        oh, ov = pl.pallas_call(
            body,
            out_shape=[jax.ShapeDtypeStruct((4 * SEGS, FAR * G, N), jnp.bfloat16), pltpu.VMEM((4 * SEGS, NEAR * G, N), jnp.bfloat16)],
            in_specs=[pl.BlockSpec(memory_space=pl.ANY)],
            out_specs=[pl.BlockSpec(memory_space=pl.ANY), pl.BlockSpec(memory_space=pltpu.VMEM)],
            scratch_shapes=[
                pltpu.VMEM((2, NI, R, N), jnp.float32),
                pltpu.VMEM((NS, 8, SLOT * LANES), jnp.int32),
                pltpu.VMEM((NY, 8, SLOT * LANES), jnp.int32),
                pltpu.VMEM((NX, 8, SLOT * LANES), jnp.int32),
                pltpu.VMEM((REACH, 8, LANES), jnp.int32),
                pltpu.VMEM((3, 8, LANES), jnp.int32),
                pltpu.VMEM((3, 8, N), jnp.int32),
                pltpu.SMEM((3, max(NS, NY, NX)), jnp.int32),
                DMA((2, NI)), DMA((4, PER, 2)), DMA((P + 1, NS)), DMA((P + 1, NY)), DMA((P + 1, NY)), DMA((P + 1, NX)),
                REG((NY,)), REG((NX,)),
            ],
            compiler_params=pltpu.CompilerParams(collective_id=0, **cp),
        )(x)
        def tiles(o):
            a, r, n = o.shape
            return o.reshape(a, r // 8, 8, n // 128, 128).transpose(0, 1, 3, 2, 4).reshape(a, r * n // 1024, 8, 128)
        out = jnp.concatenate([tiles(oh), tiles(ov)], axis=1)
        return out.reshape(2 * M // 8, N // 128, 8, 128).transpose(0, 2, 1, 3).reshape(2 * M, N)
    return fn


def pallas_dist_ag_xy_y_m65536_n1024_kernel(x):
    return make(order="p f y f r o f x f")(x)
```

```python
import contextlib

import jax
import jax.numpy as jnp
import numpy as np
from jax import lax
from jax.experimental import pallas as pl
from jax.experimental.pallas import tpu as pltpu

LANES = 256
GROUPS = 8
RATE = 27
CARRY = 6


def _i32(v):
    return np.uint32(v).view(np.int32)


def _bytes(v):
    return _i32(v * 0x01010101)


def _shl(x, n):
    return lax.shift_left(x, jnp.full_like(x, n) if isinstance(n, int) else n)


def _shr(x, n):
    return lax.shift_right_logical(x, jnp.full_like(x, n) if isinstance(n, int) else n)


def _is_short(c):
    return c % 4 == 0


def _first_bit(c):
    return (RATE * c) % 4 * 8


def _sign_mantissa(a, b):
    low = (a & _i32(0x007F007F)) | (_shr(a, 8) & _i32(0x00800080))
    high = (_shl(b, 8) & _i32(0x7F007F00)) | (b & _i32(0x80008000))
    return low | high


def _exponents(a, b):
    return (_shr(a, 7) & _i32(0x00FF00FF)) | (_shl(b, 1) & _i32(0xFF00FF00))


def _join(sm, e):
    a = (sm & _i32(0x007F007F)) | (_shl(sm, 8) & _i32(0x80008000))
    b = (_shr(sm, 8) & _i32(0x007F007F)) | (sm & _i32(0x80008000))
    return a | (_shl(e, 7) & _i32(0x7F807F80)), b | (_shr(e, 1) & _i32(0x7F807F80))


def _rank(d):
    ge16 = _shr(d + _bytes(128 - 16), 7) & _bytes(1)
    d = ((d + _bytes(15) + ge16) & _bytes(15)) | (d & _bytes(48))
    ge1 = _shr(d + _bytes(128 - 1), 7) & _bytes(1)
    ge5 = _shr(d + _bytes(128 - 5), 7) & _bytes(1)
    return d + _bytes(4) + ge5 - (_shl(ge1, 2) + ge1)


def _unrank(r):
    ge4 = (r + _bytes(128 - 4)) & _bytes(128)
    ge5 = (r + _bytes(128 - 5)) & _bytes(128)
    d = r + _bytes(1) + _shr(ge5, 5) - (_shr(ge4, 5) + _shr(ge4, 7))
    lt16 = _shr(_bytes(128 + 15) - d, 7) & _bytes(1)
    return ((d + lt16) & _bytes(15)) | (d & _bytes(48))


def _encode(exps, base, carry, end, c):
    plain = seen = None
    unary = []
    for i, e in enumerate(exps):
        d = base - e
        seen = d if seen is None else seen | d
        r = _rank(d)
        bit = _shl(r & _bytes(1), i) if i else r & _bytes(1)
        plain = bit if plain is None else plain | bit
        unary.append(_shr(r, 1) & _bytes(31))

    strings = []
    longest = None
    for half in range(2):
        lo = hi = total = None
        for z in reversed(unary[4 * half : 4 * half + 4]):
            n = z + _shr(z, 16)
            n = ((n + _shr(n, 8)) & 0xFF) + 4
            longest = n if longest is None else jnp.maximum(longest, n)
            total = n if total is None else total + n
            if lo is not None:
                spilled = _shr(lo, (32 - n) & 31)
                hi = spilled if hi is None else _shl(hi, n & 31) | spilled
            for k in reversed(range(4)):
                lo = jnp.ones_like(z) if lo is None else _shl(lo, 1) | 1
                lo = _shl(lo, (_shr(z, 8 * k) if k else z) & 31)
        longest = jnp.maximum(longest, _shr(total, 1))
        strings.append((lo, hi, total))
    misfit = (seen & _bytes(0xC0)) | _shr(longest, 5)

    words = list(carry) + [None] * 7
    bad = None
    for g in range(GROUPS):
        block = slice(g // 2 * LANES, (g // 2 + 1) * LANES)
        lo, hi, total = (v[:, block] for v in strings[g % 2])
        first = RATE * g // 32
        start = jnp.maximum(end, _first_bit(c) + RATE * g)
        end = start + total
        skip = _shr(start, 5) - first
        far = _shr(skip, 3) if g % 2 else _shr(skip, 3) | misfit[:, block]
        bad = far if bad is None else bad | far
        s = start & 31
        back = s ^ 31
        pieces = [_shl(lo, s), _shr(_shr(lo, 1), back) | _shl(hi, s), _shr(_shr(hi, 1), back)]
        for d in (1, 2, 4):
            move = (skip & d) != 0
            pieces = [
                jnp.where(move, pieces[i - d] if i >= d else 0, pieces[i] if i < len(pieces) else 0)
                for i in range(min(len(pieces) + d, len(words) - first))
            ]
        for i, p in enumerate(pieces, first):
            words[i] = p if words[i] is None else words[i] | p
    return plain, words, end, bad


def _decode(plain, words, base, end, c):
    unary = [[None] * GROUPS for _ in range(4)]
    for g in range(GROUPS):
        first = RATE * g // 32
        start = jnp.maximum(end, _first_bit(c) + RATE * g)
        skip = _shr(start, 5) - first
        pieces = words[first : first + 10]
        for d in (4, 2, 1):
            move = (skip & d) != 0
            pieces = [
                jnp.where(move, pieces[i + d], p) if i + d < len(pieces) else p
                for i, p in enumerate(pieces[: d + 2])
            ]
        s = start & 31
        back = s ^ 31
        lo = _shr(pieces[0], s) | _shl(_shl(pieces[1], 1), back)
        hi = _shr(pieces[1], s) | _shl(_shl(pieces[2], 1), back)
        end = start
        for q in range(4):
            rest, ones = lo, None
            for k in range(4):
                cleared = rest & (rest - 1)
                one = pltpu.bitcast((rest ^ cleared).astype(jnp.float32), jnp.int32)
                one = _shr(one, 23 - 8 * k) if k < 3 else _shl(one, 1)
                rest, ones = cleared, one if ones is None else ones | one
            unary[q][g] = ones - _shl(ones, 8) - _i32(0x0101017F)
            n = _shr(ones, 24) - 126
            end = end + n
            if q < 3:
                lo = _shr(lo, n) | _shl(hi, 32 - n)
            if q < 2:
                hi = _shr(hi, n)
    exps = []
    for i in range(8):
        z = jnp.concatenate(unary[i % 4][i // 4 :: 2], axis=1)
        bit = (_shr(plain, i) if i else plain) & _bytes(1)
        exps.append(base - _unrank(_shl(z, 1) | bit))
    return exps, end


PIECE = 128
FAR, NEAR = 9, 7
LOADS, SENDS, RECVS = 3, 2, 4

PLAIN, SIGNMAN, TAIL, VERBATIM, END = 7, 11, 23, 43, 75


def make(scopes=False, **params):
    def kernel(x_ref, far_ref, near_ref, in_buf, send_buf, y_buf, x_buf, carry_ref, end_ref,
               base_ref, verbatim_ref, in_sem, out_sem, y_send, y_recv, x_send, x_recv,
               y_free, x_free):
        shard, n = x_ref.shape
        pieces = shard // 2 // PIECE
        chunks = pieces // 2
        far_chunks = pieces // (FAR + NEAR) * FAR // 2
        wide = n // LANES

        my_x, my_y = lax.axis_index("x"), lax.axis_index("y")
        y_peer, x_peer = (my_x, 1 - my_y), (1 - my_x, my_y)
        SENT, KEPT, FROM_Y, FROM_X = range(4)
        half = (my_x, 1 - my_x, my_x, 1 - my_x)
        shard_of = (my_y, my_y, 1 - my_y, 1 - my_y)

        def rows(i):
            return pl.ds(pl.multiple_of(i * PIECE, PIECE), PIECE)

        def blocks(first, count=1):
            return pl.ds(first * LANES, count * LANES)

        def load(s, c, i):
            u = 2 * c + i
            v = jnp.maximum(u - 2 * far_chunks, 0)
            piece = jnp.where(
                c < far_chunks,
                u // FAR * (FAR + NEAR) + u % FAR,
                v // NEAR * (FAR + NEAR) + FAR + v % NEAR,
            )
            return pltpu.make_async_copy(
                x_ref.at[rows(half[s] * pieces + piece)],
                in_buf.at[s, c % LOADS, rows(i)],
                in_sem.at[s, c % LOADS, i],
            )

        def result(s, c, i):
            v = 2 * (jnp.where(c < far_chunks, chunks - 2 + c % 2, c) - far_chunks) + i
            first = (2 * shard_of[s] + half[s]) * (pieces // (FAR + NEAR))
            return near_ref.at[first + v // NEAR, rows(v % NEAR)]

        def store(s, c, i):
            u = 2 * c + i
            first = (2 * shard_of[s] + half[s]) * (pieces // (FAR + NEAR))
            return pltpu.make_async_copy(
                result(s, c, i), far_ref.at[first + u // FAR, rows(u % FAR)], out_sem.at[s, c % 2, i]
            )

        def before_result(s, c):
            @pl.when((c >= 2) & (c < far_chunks + 2))
            def _():
                for i in range(2):
                    store(s, c - 2, i).wait()

        def after_result(s, c):
            @pl.when(c < far_chunks)
            def _():
                for i in range(2):
                    store(s, c, i).start()

        def put(s, c, values):
            dst = [result(s, c, i) for i in range(2)]
            for k, v in enumerate(values):
                dst[k // 8][pl.ds(16 * (k % 8), 16), :] = v

        def to_y(c, lo, hi, part):
            slot, far_slot = c % SENDS, c % RECVS
            return pltpu.make_async_remote_copy(
                send_buf.at[slot, :, blocks(lo, hi - lo)],
                y_buf.at[far_slot, :, blocks(lo, hi - lo)],
                y_send.at[int(lo >= VERBATIM), slot],
                y_recv.at[part, far_slot],
                device_id=y_peer,
                device_id_type=pl.DeviceIdType.MESH,
            )

        def to_x(c, lo, hi):
            slot = c % RECVS
            return pltpu.make_async_remote_copy(
                y_buf.at[slot, :, blocks(lo, hi - lo)],
                x_buf.at[slot, :, blocks(lo, hi - lo)],
                x_send.at[int(lo >= VERBATIM), slot],
                x_recv.at[int(lo >= TAIL) + int(lo >= VERBATIM), slot],
                device_id=x_peer,
                device_id_type=pl.DeviceIdType.MESH,
            )

        def from_start(c, fn):
            pl.when(_is_short(c))(lambda: fn(1))
            pl.when(jnp.logical_not(_is_short(c)))(lambda: fn(0))

        def anywhere(mask):
            return jnp.max(jnp.where(mask, 1, 0))

        def is_verbatim(buf, c):
            slot = c % RECVS
            last = jnp.where(_is_short(c), buf[slot, :, blocks(1)], buf[slot, :, blocks(0)])
            return anywhere(last == 0)

        def rounded(s, c, k):
            return in_buf[s, c % LOADS, pl.ds(16 * k, 16), :].astype(jnp.bfloat16)

        def pack(c):
            slot = c % SENDS

            @pl.when(c >= SENDS)
            def _():
                from_start(c - SENDS, lambda lo: to_y(c - SENDS, lo, VERBATIM, 0).wait_send())
                pl.when(verbatim_ref[0, slot] != 0)(lambda: to_y(c - SENDS, VERBATIM, END, 0).wait_send())

            @pl.when(c < chunks)
            def _():
                early = (TAIL - SIGNMAN) // wide
                load(SENT, c, 0).wait()
                for i in range(early):
                    a, b = (pltpu.bitcast(rounded(SENT, c, k), jnp.int32) for k in (2 * i, 2 * i + 1))
                    send_buf[slot, :, blocks(SIGNMAN + wide * i, wide)] = _sign_mantissa(a, b)
                pl.when(c == 0)(lambda: pl.semaphore_wait(barrier, 2))
                pl.when(c >= RECVS)(lambda: pl.semaphore_wait(y_free.at[c % RECVS], 1))
                to_y(c, SIGNMAN, TAIL, 0).start()

                @pl.when(c == 0)
                def _():
                    w = pltpu.bitcast(rounded(SENT, c, 0), jnp.int32)
                    total = jnp.sum((_shr(w, 7) & 0xFF) + (_shr(w, 23) & 0xFF))
                    mean = (total + 16 * n * 15 // 16) // (16 * n)
                    base = jnp.full_like(w, jnp.clip(mean + 3, 64, 255))
                    carry_ref[0] = base[:, :LANES]
                    for i in range(1, CARRY):
                        carry_ref[i] = jnp.zeros((8, LANES), jnp.int32)
                    start_stream(0, base)

                load(SENT, c, 1).wait()
                before_result(SENT, c)
                values = [rounded(SENT, c, k) for k in range(16)]
                put(SENT, c, values)
                words = [pltpu.bitcast(v, jnp.int32) for v in values]
                pairs = list(zip(words[0::2], words[1::2]))
                for i in range(early, 8):
                    send_buf[slot, :, blocks(SIGNMAN + wide * i, wide)] = _sign_mantissa(*pairs[i])
                carry = [carry_ref[i] for i in range(CARRY)]
                plain, stream, end, bad = _encode(
                    [_exponents(*p) for p in pairs], base_ref[0], carry, end_ref[0], c
                )
                send_buf[slot, :, blocks(PLAIN, wide)] = plain
                for i in range(7):
                    send_buf[slot, :, blocks(6 - i)] = stream[i]
                short = _is_short(c)
                for i in range(CARRY):
                    carry_ref[i] = jnp.where(short, stream[6 + i], stream[7 + i])
                end = jnp.maximum(end - jnp.where(short, 6 * 32, 7 * 32), 0)
                end_ref[0] = end
                room = jnp.where(_is_short(c + 1), 5 * 32, 6 * 32)
                last = jnp.where(short, stream[5], stream[6])
                verbatim = anywhere((bad != 0) | (end > room) | (last == 0))
                verbatim_ref[0, slot] = verbatim

                @pl.when(verbatim != 0)
                def _():
                    zero = jnp.zeros((8, LANES), jnp.int32)
                    send_buf[slot, :, blocks(0)] = zero
                    for i in range(CARRY):
                        send_buf[slot, :, blocks(6 - i)] = carry[i]
                        carry_ref[i] = zero
                    end_ref[0] = zero
                    for i in range(8):
                        a, b = (pltpu.bitcast(rounded(SENT, c, k), jnp.int32) for k in (2 * i, 2 * i + 1))
                        send_buf[slot, :, blocks(VERBATIM + wide * i, wide)] = _exponents(a, b)

                from_start(c, lambda lo: to_y(c, lo, SIGNMAN, 1).start())
                to_y(c, TAIL, (TAIL + VERBATIM) // 2, 2).start()
                to_y(c, (TAIL + VERBATIM) // 2, VERBATIM, 3).start()
                pl.when(verbatim != 0)(lambda: to_y(c, VERBATIM, END, 4).start())
                after_result(SENT, c)
                prefetch(SENT, c)

            @pl.when(c == chunks)
            def _():
                for i in range(CARRY - 1):
                    send_buf[slot, :, blocks(6 - i)] = carry_ref[i]
                pl.semaphore_wait(y_free.at[chunks % RECVS], 1)
                to_y(chunks, 2, PLAIN, 1).start()

        def prefetch(s, c):
            @pl.when(c + LOADS < chunks)
            def _():
                for i in range(2):
                    load(s, c + LOADS, i).start()

        def keep(c):
            @pl.when((c >= 0) & (c < chunks))
            def _():
                for i in range(2):
                    load(KEPT, c, i).wait()
                before_result(KEPT, c)
                for i in range(2):
                    result(KEPT, c, i)[...] = in_buf[KEPT, c % LOADS, rows(i)].astype(jnp.bfloat16)
                after_result(KEPT, c)
                prefetch(KEPT, c)

        def pass_on(c, part):
            def blocks_on(lo, hi, k=part):
                to_y(c, lo, hi, k).wait_recv()
                to_x(c, lo, hi).start()

            @pl.when((c >= 0) & (c < chunks))
            def _():
                if part == 0:
                    pl.when(c >= RECVS)(lambda: pl.semaphore_wait(x_free.at[c % RECVS], 1))
                    blocks_on(SIGNMAN, TAIL)
                elif part == 1:
                    from_start(c, lambda lo: blocks_on(lo, SIGNMAN))
                    verbatim_ref[1, c % RECVS] = is_verbatim(y_buf, c)
                elif part == 2:
                    blocks_on(TAIL, (TAIL + VERBATIM) // 2)
                else:
                    blocks_on((TAIL + VERBATIM) // 2, VERBATIM)
                    pl.when(verbatim_ref[1, c % RECVS] != 0)(lambda: blocks_on(VERBATIM, END, 4))

            if part == 1:

                @pl.when(c == chunks)
                def _():
                    pl.semaphore_wait(x_free.at[chunks % RECVS], 1)
                    blocks_on(2, PLAIN)

        def start_stream(k, base):
            end_ref[k] = jnp.full((8, LANES), 8, jnp.int32)
            base = base | _shl(base, 8)
            base_ref[k] = base | _shl(base, 16)

        def unpack(s, buf, c):
            k, slot = s - 1, c % RECVS

            @pl.when(c == 0)
            def _():
                base = buf[0, :, blocks(6)] & 0xFF
                start_stream(k, jnp.concatenate([base] * wide, axis=1))

            def finish(exps):
                words = []
                for i, e in enumerate(exps):
                    words += _join(buf[slot, :, blocks(SIGNMAN + wide * i, wide)], e)
                put(s, c, [pltpu.bitcast(w, jnp.bfloat16) for w in words])

            before_result(s, c)
            verbatim = verbatim_ref[k, slot]

            @pl.when(verbatim == 0)
            def _():
                short = _is_short(c)
                mine = [buf[slot, :, blocks(6 - i)] for i in range(7)]
                later = [buf[(c + 1) % RECVS, :, blocks(6 - i)] for i in range(CARRY)]
                stream = mine[:6] + [jnp.where(short, a, b) for a, b in zip(later, mine[6:] + later)]
                exps, end = _decode(
                    buf[slot, :, blocks(PLAIN, wide)], stream + later[-1:], base_ref[k], end_ref[k], c
                )
                end_ref[k] = jnp.maximum(end - jnp.where(short, 6 * 32, 7 * 32), 0)
                finish(exps)

            @pl.when(verbatim != 0)
            def _():
                end_ref[k] = jnp.zeros((8, LANES), jnp.int32)
                finish([buf[slot, :, blocks(VERBATIM + wide * i, wide)] for i in range(8)])

            after_result(s, c)

        def unpack_y(c):
            pl.when((c >= 0) & (c < chunks))(lambda: unpack(FROM_Y, y_buf, c))

        def free_y(c):
            @pl.when((c >= 0) & (c < chunks))
            def _():
                from_start(c, lambda lo: to_x(c, lo, VERBATIM).wait_send())
                pl.when(verbatim_ref[1, c % RECVS] != 0)(lambda: to_x(c, VERBATIM, END).wait_send())

                @pl.when(c + RECVS <= chunks)
                def _():
                    pl.semaphore_signal(y_free.at[c % RECVS], 1, device_id=y_peer,
                                        device_id_type=pl.DeviceIdType.MESH)

        def unpack_x(c):
            @pl.when((c >= 0) & (c < chunks))
            def _():
                to_x(c, TAIL, VERBATIM).wait_recv()
                pl.when(verbatim_ref[2, c % RECVS] != 0)(lambda: to_x(c, VERBATIM, END).wait_recv())

            @pl.when((c >= -1) & (c + 1 < chunks))
            def _():
                from_start(c + 1, lambda lo: to_x(c + 1, lo, TAIL).wait_recv())
                verbatim_ref[2, (c + 1) % RECVS] = is_verbatim(x_buf, c + 1)

            pl.when(c + 1 == chunks)(lambda: to_x(chunks, 2, PLAIN).wait_recv())

            @pl.when((c >= 0) & (c < chunks))
            def _():
                unpack(FROM_X, x_buf, c)

                @pl.when(c + RECVS <= chunks)
                def _():
                    pl.semaphore_signal(x_free.at[c % RECVS], 1, device_id=x_peer,
                                        device_id_type=pl.DeviceIdType.MESH)

        for c in range(LOADS + 1):
            for s, k in ((SENT, c), (KEPT, c - 1)):
                if 0 <= k < LOADS:
                    for i in range(2):
                        load(s, k, i).start()
        for slot in range(RECVS):
            y_buf[slot, :, blocks(0)] = jnp.zeros((8, LANES), jnp.int32)
            x_buf[slot, :, blocks(0)] = jnp.zeros((8, LANES), jnp.int32)
        barrier = pltpu.get_barrier_semaphore()
        for peer in (y_peer, x_peer):
            pl.semaphore_signal(barrier, 1, device_id=peer, device_id_type=pl.DeviceIdType.MESH)

        def step(t, _):
            for name, work in (
                ("f0", lambda: pass_on(t - 1, 0)),
                ("p", lambda: pack(t)),
                ("f1", lambda: pass_on(t - 1, 1)),
                ("y", lambda: unpack_y(t - 2)),
                ("f2", lambda: pass_on(t - 1, 2)),
                ("r", lambda: free_y(t - 2)),
                ("o", lambda: keep(t - 1)),
                ("f3", lambda: pass_on(t - 1, 3)),
                ("x", lambda: unpack_x(t - 2)),
            ):
                with jax.named_scope(name) if scopes else contextlib.nullcontext():
                    work()

        lax.fori_loop(0, chunks + 2, step, None)
        to_y(chunks, 2, PLAIN, 1).wait_send()
        to_x(chunks, 2, PLAIN).wait_send()

    def fn(x):
        shard, n = x.shape
        segments = 2 * shard // (PIECE * (FAR + NEAR))
        dma, regular = pltpu.SemaphoreType.DMA, pltpu.SemaphoreType.REGULAR
        message = (8, END * LANES)
        far, near = pl.pallas_call(
            kernel,
            out_shape=[
                jax.ShapeDtypeStruct((segments, FAR * PIECE, n), jnp.bfloat16),
                pltpu.VMEM((segments, NEAR * PIECE, n), jnp.bfloat16),
            ],
            in_specs=[pl.BlockSpec(memory_space=pl.ANY)],
            out_specs=[pl.BlockSpec(memory_space=pl.ANY), pl.BlockSpec(memory_space=pltpu.VMEM)],
            scratch_shapes=[
                pltpu.VMEM((2, LOADS, 2 * PIECE, n), x.dtype),
                pltpu.VMEM((SENDS,) + message, jnp.int32),
                pltpu.VMEM((RECVS,) + message, jnp.int32),
                pltpu.VMEM((RECVS,) + message, jnp.int32),
                pltpu.VMEM((CARRY, 8, LANES), jnp.int32),
                pltpu.VMEM((3, 8, LANES), jnp.int32),
                pltpu.VMEM((3, 8, n), jnp.int32),
                pltpu.SMEM((3, RECVS), jnp.int32),
                dma((2, LOADS, 2)),
                dma((4, 2, 2)),
                dma((2, SENDS)),
                dma((5, RECVS)),
                dma((2, RECVS)),
                dma((3, RECVS)),
                regular((RECVS,)),
                regular((RECVS,)),
            ],
            compiler_params=pltpu.CompilerParams(collective_id=0, **params),
        )(x)

        def tiles(a):
            a = a.reshape(segments, -1, 8, n // 128, 128).transpose(0, 1, 3, 2, 4)
            return a.reshape(segments, -1, 8, 128)

        out = jnp.concatenate([tiles(far), tiles(near)], axis=1)
        return out.reshape(-1, n // 128, 8, 128).transpose(0, 2, 1, 3).reshape(2 * shard, n)

    return fn


def pallas_dist_ag_xy_y_m65536_n1024_kernel(x):
    return make()(x)
```

```python
import jax
import jax.numpy as jnp
import numpy as np
from jax import lax
from jax.experimental import pallas as pl
from jax.experimental.pallas import tpu as pltpu

LANES = 256
GROUPS = 8
MIN_RATE, MAX_RATE = 27, 32
SHIPPED = GROUPS * MAX_RATE // 32
WAITING = SHIPPED - 1


def _i32(v):
    return np.uint32(v).view(np.int32)


def _bytes(v):
    return _i32(v * 0x01010101)


def _shl(x, n):
    return lax.shift_left(x, jnp.full_like(x, n) if isinstance(n, int) else n)


def _shr(x, n):
    return lax.shift_right_logical(x, jnp.full_like(x, n) if isinstance(n, int) else n)


def _shipped(c, rate):
    return rate * (c + 1) // 4 - rate * c // 4


def _first_bit(c, rate):
    return rate * c % 4 * 8


def _sign_mantissa(a, b):
    low = (a & _i32(0x007F007F)) | (_shr(a, 8) & _i32(0x00800080))
    high = (_shl(b, 8) & _i32(0x7F007F00)) | (b & _i32(0x80008000))
    return low | high


def _exponents(a, b):
    return (_shr(a, 7) & _i32(0x00FF00FF)) | (_shl(b, 1) & _i32(0xFF00FF00))


def _join(sm, e):
    a = (sm & _i32(0x007F007F)) | (_shl(sm, 8) & _i32(0x80008000))
    b = (_shr(sm, 8) & _i32(0x007F007F)) | (sm & _i32(0x80008000))
    return a | (_shl(e, 7) & _i32(0x7F807F80)), b | (_shr(e, 1) & _i32(0x7F807F80))


def _rank(d):
    ge16 = _shr(d + _bytes(128 - 16), 5) & _bytes(4)
    d = ((d + _bytes(12) + ge16) & _bytes(15)) | (d & _bytes(48))
    ge1 = _shr(d + _bytes(128 - 1), 7) & _bytes(1)
    ge5 = _shr(d + _bytes(128 - 5), 7) & _bytes(1)
    return d + _bytes(4) + ge5 - (_shl(ge1, 2) + ge1)


def _unrank(r):
    ge4 = (r + _bytes(128 - 4)) & _bytes(128)
    ge5 = (r + _bytes(128 - 5)) & _bytes(128)
    d = r + _bytes(1) + _shr(ge5, 5) - (_shr(ge4, 5) + _shr(ge4, 7))
    lt16 = _shr(_bytes(128 + 15) - d, 5) & _bytes(4)
    return ((d + lt16) & _bytes(15)) | (d & _bytes(48))


def _encode(exps, base):
    plain = seen = None
    unary = []
    for i, e in enumerate(exps):
        d = base - e
        seen = d if seen is None else seen | d
        r = _rank(d)
        bit = _shl(r & _bytes(1), i) if i else r & _bytes(1)
        plain = bit if plain is None else plain | bit
        unary.append(_shr(r, 1) & _bytes(31))

    strings = []
    longest = None
    for group in (unary[:4], unary[4:]):
        lo = hi = total = None
        for z in reversed(group):
            n = z + _shr(z, 16)
            n = ((n + _shr(n, 8)) & 0xFF) + 4
            longest = n if longest is None else jnp.maximum(longest, n)
            total = n if total is None else total + n
            if lo is not None:
                spilled = _shr(lo, (32 - n) & 31)
                hi = spilled if hi is None else _shl(hi, n & 31) | spilled
            for k in reversed(range(4)):
                lo = jnp.ones_like(z) if lo is None else _shl(lo, 1) | 1
                lo = _shl(lo, (_shr(z, 8 * k) if k else z) & 31)
        longest = jnp.maximum(longest, _shr(total, 1))
        strings.append((lo, hi, total))
    return plain, strings, (seen & _bytes(0xC0)) | _shr(longest, 5)


def _append(strings, waiting, end, c, rate):
    stream = list(waiting) + [None] * SHIPPED
    behind = None
    for g in range(GROUPS):
        lo, hi, total = (v[:, g // 2 * LANES : (g // 2 + 1) * LANES] for v in strings[g % 2])
        first = MIN_RATE * g // 32
        start = jnp.maximum(end, _first_bit(c, rate) + rate * g)
        end = start + total
        skip = _shr(start, 5) - first
        behind = skip if behind is None else behind | skip
        s = start & 31
        back = s ^ 31
        parts = [_shl(lo, s), _shr(_shr(lo, 1), back) | _shl(hi, s), _shr(_shr(hi, 1), back)]
        for d in (1, 2, 4):
            move = (skip & d) != 0
            parts = [
                jnp.where(move, parts[i - d] if i >= d else 0, parts[i] if i < len(parts) else 0)
                for i in range(len(parts) + d)
            ]
        for i, p in enumerate(parts, first):
            stream[i] = p if stream[i] is None else stream[i] | p
    return stream, end, _shr(behind, 3)


def _decode(plain, stream, base, end, c, rate):
    unary = [[None] * GROUPS for _ in range(4)]
    for g in range(GROUPS):
        first = MIN_RATE * g // 32
        start = jnp.maximum(end, _first_bit(c, rate) + rate * g)
        skip = _shr(start, 5) - first
        parts = stream[first:]
        for d in (4, 2, 1):
            move = (skip & d) != 0
            parts = [jnp.where(move, parts[i + d], parts[i]) for i in range(d + 2)]
        s = start & 31
        back = s ^ 31
        lo = _shr(parts[0], s) | _shl(_shl(parts[1], 1), back)
        hi = _shr(parts[1], s) | _shl(_shl(parts[2], 1), back)
        end = start
        for q in range(4):
            rest, ones = lo, None
            for k in range(4):
                cleared = rest & (rest - 1)
                one = pltpu.bitcast((rest ^ cleared).astype(jnp.float32), jnp.int32)
                one = _shr(one, 23 - 8 * k) if k < 3 else _shl(one, 1)
                rest, ones = cleared, one if ones is None else ones | one
            unary[q][g] = ones - _shl(ones, 8) - _i32(0x0101017F)
            n = _shr(ones, 24) - 126
            end = end + n
            if q < 3:
                lo = _shr(lo, n) | _shl(hi, 32 - n)
            if q < 2:
                hi = _shr(hi, n)
    exps = []
    for i in range(8):
        z = jnp.concatenate(unary[i % 4][i // 4 :: 2], axis=1)
        bit = (_shr(plain, i) if i else plain) & _bytes(1)
        exps.append(base - _unrank(_shl(z, 1) | bit))
    return exps, end


PIECE = 128
FAR, NEAR = 9, 7
LOADS, SENDS, RECVS = 3, 2, 4

PLAIN, SIGNS, TAIL, LAST, VERBATIM, END = 8, 12, 24, 34, 44, 76

SENT, KEPT, FROM_Y, FROM_X = range(4)


def _kernel(
    x_ref, far_ref, near_ref,
    in_buf, send_buf, y_buf, x_buf, waiting_ref, end_ref, base_ref, rate_ref, verbatim_ref,
    in_sem, out_sem, y_send, y_recv, x_send, x_recv, y_free, x_free,
):
    shard, n = x_ref.shape
    pieces = shard // 2 // PIECE
    chunks = pieces // 2
    segments = pieces // (FAR + NEAR)
    far_chunks = segments * FAR // 2
    wide = n // LANES

    my_x, my_y = lax.axis_index("x"), lax.axis_index("y")
    y_peer = dict(device_id=(my_x, 1 - my_y), device_id_type=pl.DeviceIdType.MESH)
    x_peer = dict(device_id=(1 - my_x, my_y), device_id_type=pl.DeviceIdType.MESH)
    half = (my_x, 1 - my_x, my_x, 1 - my_x)
    quarter = [2 * y + h for y, h in zip((my_y, my_y, 1 - my_y, 1 - my_y), half)]

    def rows(i):
        return pl.ds(pl.multiple_of(i * PIECE, PIECE), PIECE)

    def blocks(first, count=1):
        return pl.ds(first * LANES, count * LANES)

    def zeros():
        return jnp.zeros((8, LANES), jnp.int32)

    def anywhere(mask):
        return jnp.max(jnp.where(mask, 1, 0))

    def when_chunk(c):
        return pl.when((c >= 0) & (c < chunks))


    def load(s, c, i):
        u = 2 * c + i
        v = jnp.maximum(u - 2 * far_chunks, 0)
        piece = jnp.where(
            c < far_chunks,
            u // FAR * (FAR + NEAR) + u % FAR,
            v // NEAR * (FAR + NEAR) + FAR + v % NEAR,
        )
        return pltpu.make_async_copy(
            x_ref.at[rows(half[s] * pieces + piece)],
            in_buf.at[s, c % LOADS, rows(i)],
            in_sem.at[s, c % LOADS, i],
        )

    def prefetch(s, c):
        @pl.when(c + LOADS < chunks)
        def _():
            for i in range(2):
                load(s, c + LOADS, i).start()

    def result(s, c, i):
        v = 2 * (jnp.where(c < far_chunks, chunks - 2 + c % 2, c) - far_chunks) + i
        return near_ref.at[quarter[s] * segments + v // NEAR, rows(v % NEAR)]

    def store(s, c, i):
        u = 2 * c + i
        return pltpu.make_async_copy(
            result(s, c, i),
            far_ref.at[quarter[s] * segments + u // FAR, rows(u % FAR)],
            out_sem.at[s, c % 2, i],
        )

    def before_result(s, c):
        @pl.when((c >= 2) & (c < far_chunks + 2))
        def _():
            for i in range(2):
                store(s, c - 2, i).wait()

    def after_result(s, c):
        @pl.when(c < far_chunks)
        def _():
            for i in range(2):
                store(s, c, i).start()

    def put(s, c, values):
        dst = [result(s, c, i) for i in range(2)]
        for k, v in enumerate(values):
            dst[k // 8][pl.ds(16 * (k % 8), 16), :] = v


    def to_y(c, lo, hi, part=0):
        return pltpu.make_async_remote_copy(
            send_buf.at[c % SENDS, :, blocks(lo, hi - lo)],
            y_buf.at[c % RECVS, :, blocks(lo, hi - lo)],
            y_send.at[int(lo >= VERBATIM), c % SENDS],
            y_recv.at[part, c % RECVS],
            **y_peer,
        )

    def to_x(c, lo, hi):
        return pltpu.make_async_remote_copy(
            y_buf.at[c % RECVS, :, blocks(lo, hi - lo)],
            x_buf.at[c % RECVS, :, blocks(lo, hi - lo)],
            x_send.at[int(lo >= VERBATIM), c % RECVS],
            x_recv.at[int(lo >= TAIL) + int(lo >= VERBATIM), c % RECVS],
            **x_peer,
        )

    def from_start(s, c, fn):
        start = jnp.where(c == 0, 0, SHIPPED - _shipped(c, rate_ref[s]))
        for lo in range(3):
            pl.when(start == lo)(lambda: fn(lo))

    def by_shipped(count, choices):
        fewer = jnp.where(count == SHIPPED - 1, choices[1], choices[2])
        return jnp.where(count == SHIPPED, choices[0], fewer)

    def begin(s, base):
        end_ref[s] = zeros() + 16
        base = base | _shl(base, 8)
        base_ref[s] = base | _shl(base, 16)

    def read_head(s, buf, c):
        slot = c % RECVS

        @pl.when(c == 0)
        def _():
            head = buf[0, :, blocks(SHIPPED - 1)]
            begin(s, jnp.concatenate([head & 0xFF] * wide, axis=1))
            rate_ref[s] = jnp.max(_shr(head, 8) & 0xFF)

        first = by_shipped(_shipped(c, rate_ref[s]), [buf[slot, :, blocks(i)] for i in range(3)])
        verbatim_ref[s, slot] = anywhere(first == 0)


    def pack(c):
        slot = c % SENDS

        def rounded(k):
            return in_buf[SENT, c % LOADS, pl.ds(16 * k, 16), :].astype(jnp.bfloat16)

        def pair(i):
            return [pltpu.bitcast(rounded(k), jnp.int32) for k in (2 * i, 2 * i + 1)]

        @pl.when(c >= SENDS)
        def _():
            sent = c - SENDS
            from_start(SENT, sent, lambda lo: to_y(sent, lo, VERBATIM).wait_send())
            pl.when(verbatim_ref[SENT, slot] != 0)(lambda: to_y(sent, VERBATIM, END).wait_send())

        @when_chunk(c)
        def _():
            early = (TAIL - SIGNS) // wide
            load(SENT, c, 0).wait()
            for i in range(early):
                send_buf[slot, :, blocks(SIGNS + wide * i, wide)] = _sign_mantissa(*pair(i))
            pl.when(c == 0)(lambda: pl.semaphore_wait(barrier, 2))
            pl.when(c >= RECVS)(lambda: pl.semaphore_wait(y_free.at[c % RECVS], 1))
            to_y(c, SIGNS, TAIL, 0).start()

            @pl.when(c == 0)
            def _():
                e = _exponents(*pair(0))
                total = jnp.sum((e & 0xFF) + _shr(e, 24))
                mean = (total + 15 * n) // (16 * n)
                begin(SENT, jnp.full_like(e, jnp.clip(mean + 6, 64, 255)))

            load(SENT, c, 1).wait()
            before_result(SENT, c)
            values = [rounded(k) for k in range(16)]
            put(SENT, c, values)
            words = [pltpu.bitcast(v, jnp.int32) for v in values]
            pairs = list(zip(words[0::2], words[1::2]))
            for i in range(early, 8):
                send_buf[slot, :, blocks(SIGNS + wide * i, wide)] = _sign_mantissa(*pairs[i])
            plain, strings, misfit = _encode([_exponents(*p) for p in pairs], base_ref[SENT])
            send_buf[slot, :, blocks(PLAIN, wide)] = plain

            total = jnp.sum(strings[0][2] + strings[1][2])
            fitting = jnp.clip((total + 26 * n - 1) // (16 * n), MIN_RATE, MAX_RATE)
            rate = jnp.where(c == 0, fitting, rate_ref[SENT])
            rate_ref[SENT] = rate
            waiting = [waiting_ref[i] for i in range(WAITING)]
            head = (base_ref[SENT, :, blocks(0)] & 0xFF) | (rate * 256)
            waiting[0] = jnp.where(c == 0, head, waiting[0])

            stream, end, bad = _append(strings, waiting, end_ref[SENT], c, rate)
            count = _shipped(c, rate)
            for i in range(SHIPPED):
                send_buf[slot, :, blocks(SHIPPED - 1 - i)] = stream[i]
            for i in range(WAITING):
                waiting_ref[i] = by_shipped(count, [stream[SHIPPED - k + i] for k in range(3)])
            end = jnp.maximum(end - 32 * count, 0)
            end_ref[SENT] = end
            room = 32 * (_shipped(c + 1, rate) - 1)
            first = by_shipped(count, [stream[SHIPPED - 1 - k] for k in range(3)])
            for i in range(wide):
                bad = bad | misfit[:, i * LANES : (i + 1) * LANES]
            verbatim = anywhere((bad != 0) | (end > room) | (first == 0))
            verbatim_ref[SENT, slot] = verbatim

            @pl.when(verbatim != 0)
            def _():
                send_buf[slot, :, blocks(0)] = zeros()
                for i in range(WAITING):
                    send_buf[slot, :, blocks(SHIPPED - 1 - i)] = waiting[i]
                    waiting_ref[i] = zeros()
                end_ref[SENT] = zeros()
                for i in range(8):
                    send_buf[slot, :, blocks(VERBATIM + wide * i, wide)] = _exponents(*pair(i))

            from_start(SENT, c, lambda lo: to_y(c, lo, SIGNS, 1).start())
            to_y(c, TAIL, LAST, 2).start()
            to_y(c, LAST, VERBATIM, 3).start()
            pl.when(verbatim != 0)(lambda: to_y(c, VERBATIM, END, 4).start())
            after_result(SENT, c)
            prefetch(SENT, c)

        @pl.when(c == chunks)
        def _():
            for i in range(WAITING):
                send_buf[slot, :, blocks(SHIPPED - 1 - i)] = waiting_ref[i]
            pl.semaphore_wait(y_free.at[c % RECVS], 1)
            from_start(SENT, c, lambda lo: to_y(c, lo + 1, PLAIN, 1).start())

    def keep(c):
        @when_chunk(c)
        def _():
            for i in range(2):
                load(KEPT, c, i).wait()
            before_result(KEPT, c)
            for i in range(2):
                result(KEPT, c, i)[...] = in_buf[KEPT, c % LOADS, rows(i)].astype(jnp.bfloat16)
            after_result(KEPT, c)
            prefetch(KEPT, c)

    def pass_on(c, part):
        def one(lo, hi, part):
            to_y(c, lo, hi, part).wait_recv()
            to_x(c, lo, hi).start()

        @when_chunk(c)
        def _():
            if part == 0:
                pl.when(c >= RECVS)(lambda: pl.semaphore_wait(x_free.at[c % RECVS], 1))
                one(SIGNS, TAIL, 0)
            elif part == 1:
                from_start(FROM_Y, c, lambda lo: one(lo, SIGNS, 1))
                read_head(FROM_Y, y_buf, c)
            elif part == 2:
                one(TAIL, LAST, 2)
            else:
                one(LAST, VERBATIM, 3)
                pl.when(verbatim_ref[FROM_Y, c % RECVS] != 0)(lambda: one(VERBATIM, END, 4))

        if part == 1:

            @pl.when(c == chunks)
            def _():
                pl.semaphore_wait(x_free.at[c % RECVS], 1)
                from_start(FROM_Y, c, lambda lo: one(lo + 1, PLAIN, 1))

    def unpack(s, buf, c):
        slot = c % RECVS

        def finish(exps):
            words = []
            for i, e in enumerate(exps):
                words += _join(buf[slot, :, blocks(SIGNS + wide * i, wide)], e)
            put(s, c, [pltpu.bitcast(w, jnp.bfloat16) for w in words])

        before_result(s, c)
        verbatim = verbatim_ref[s, slot]

        @pl.when(verbatim == 0)
        def _():
            rate = rate_ref[s]
            count = _shipped(c, rate)
            mine = [buf[slot, :, blocks(SHIPPED - 1 - i)] for i in range(SHIPPED)]
            later = [buf[(c + 1) % RECVS, :, blocks(SHIPPED - 1 - i)] for i in range(WAITING)]
            joined = [mine[: SHIPPED - k] + later + later[:k] for k in range(3)]
            stream = mine[: SHIPPED - 2] + [
                by_shipped(count, choices) for choices in list(zip(*joined))[SHIPPED - 2 :]
            ]
            plain = buf[slot, :, blocks(PLAIN, wide)]
            exps, end = _decode(plain, stream, base_ref[s], end_ref[s], c, rate)
            end_ref[s] = jnp.maximum(end - 32 * count, 0)
            finish(exps)

        @pl.when(verbatim != 0)
        def _():
            end_ref[s] = zeros()
            finish([buf[slot, :, blocks(VERBATIM + wide * i, wide)] for i in range(8)])

        after_result(s, c)

    def receive_y(c):
        when_chunk(c)(lambda: unpack(FROM_Y, y_buf, c))

    def free_y(c):
        @when_chunk(c)
        def _():
            slot = c % RECVS
            from_start(FROM_Y, c, lambda lo: to_x(c, lo, VERBATIM).wait_send())
            pl.when(verbatim_ref[FROM_Y, slot] != 0)(lambda: to_x(c, VERBATIM, END).wait_send())
            pl.when(c + RECVS <= chunks)(lambda: pl.semaphore_signal(y_free.at[slot], 1, **y_peer))

    def receive_x(c):
        @when_chunk(c)
        def _():
            to_x(c, TAIL, VERBATIM).wait_recv()
            verbatim = verbatim_ref[FROM_X, c % RECVS]
            pl.when(verbatim != 0)(lambda: to_x(c, VERBATIM, END).wait_recv())

        @when_chunk(c + 1)
        def _():
            from_start(FROM_X, c + 1, lambda lo: to_x(c + 1, lo, TAIL).wait_recv())
            read_head(FROM_X, x_buf, c + 1)

        @pl.when(c + 1 == chunks)
        def _():
            from_start(FROM_X, c + 1, lambda lo: to_x(c + 1, lo + 1, PLAIN).wait_recv())

        @when_chunk(c)
        def _():
            slot = c % RECVS
            unpack(FROM_X, x_buf, c)
            pl.when(c + RECVS <= chunks)(lambda: pl.semaphore_signal(x_free.at[slot], 1, **x_peer))


    for c in range(LOADS + 1):
        for s, k in ((SENT, c), (KEPT, c - 1)):
            if 0 <= k < LOADS:
                for i in range(2):
                    load(s, k, i).start()
    for s in range(4):
        rate_ref[s] = MIN_RATE
    for i in range(WAITING):
        waiting_ref[i] = zeros()
    for buf in (y_buf, x_buf):
        for slot in range(RECVS):
            for i in range(2):
                buf[slot, :, blocks(i)] = zeros()
    barrier = pltpu.get_barrier_semaphore()
    pl.semaphore_signal(barrier, 1, **y_peer)
    pl.semaphore_signal(barrier, 1, **x_peer)

    def step(t, _):
        pass_on(t - 1, 0)
        pack(t)
        pass_on(t - 1, 1)
        receive_y(t - 2)
        pass_on(t - 1, 2)
        free_y(t - 2)
        keep(t - 1)
        pass_on(t - 1, 3)
        receive_x(t - 2)

    lax.fori_loop(0, chunks + 2, step, None)
    from_start(SENT, chunks, lambda lo: to_y(chunks, lo + 1, PLAIN).wait_send())
    from_start(FROM_Y, chunks, lambda lo: to_x(chunks, lo + 1, PLAIN).wait_send())


def pallas_dist_ag_xy_y_m65536_n1024_kernel(x: jax.Array):
    shard, n = x.shape
    segments = 2 * shard // (PIECE * (FAR + NEAR))
    dma, regular = pltpu.SemaphoreType.DMA, pltpu.SemaphoreType.REGULAR
    far, near = pl.pallas_call(
        _kernel,
        out_shape=[
            jax.ShapeDtypeStruct((segments, FAR * PIECE, n), jnp.bfloat16),
            pltpu.VMEM((segments, NEAR * PIECE, n), jnp.bfloat16),
        ],
        in_specs=[pl.BlockSpec(memory_space=pl.ANY)],
        out_specs=[pl.BlockSpec(memory_space=pl.ANY), pl.BlockSpec(memory_space=pltpu.VMEM)],
        scratch_shapes=[
            pltpu.VMEM((2, LOADS, 2 * PIECE, n), x.dtype),
            pltpu.VMEM((SENDS, 8, END * LANES), jnp.int32),
            pltpu.VMEM((RECVS, 8, END * LANES), jnp.int32),
            pltpu.VMEM((RECVS, 8, END * LANES), jnp.int32),
            pltpu.VMEM((WAITING, 8, LANES), jnp.int32),
            pltpu.VMEM((4, 8, LANES), jnp.int32),
            pltpu.VMEM((4, 8, n), jnp.int32),
            pltpu.SMEM((4,), jnp.int32),
            pltpu.SMEM((4, RECVS), jnp.int32),
            dma((2, LOADS, 2)),
            dma((4, 2, 2)),
            dma((2, SENDS)),
            dma((5, RECVS)),
            dma((2, RECVS)),
            dma((3, RECVS)),
            regular((RECVS,)),
            regular((RECVS,)),
        ],
        compiler_params=pltpu.CompilerParams(collective_id=0),
    )(x)

    def tiles(a):
        a = a.reshape(segments, -1, 8, n // 128, 128).transpose(0, 1, 3, 2, 4)
        return a.reshape(segments, -1, 8, 128)

    out = jnp.concatenate([tiles(far), tiles(near)], axis=1)
    return out.reshape(-1, n // 128, 8, 128).transpose(0, 2, 1, 3).reshape(2 * shard, n)
```

```python
import jax
import jax.numpy as jnp
import numpy as np
from jax import lax
from jax.experimental import pallas as pl
from jax.experimental.pallas import tpu as pltpu

LANES = 256
GROUPS = 8
MIN_RATE, MAX_RATE = 27, 32
SHIPPED = GROUPS * MAX_RATE // 32
WAITING = SHIPPED - 1


def _i32(v):
    return np.uint32(v).view(np.int32)


def _bytes(v):
    return _i32(v * 0x01010101)


def _shl(x, n):
    return lax.shift_left(x, jnp.full_like(x, n) if isinstance(n, int) else n)


def _shr(x, n):
    return lax.shift_right_logical(x, jnp.full_like(x, n) if isinstance(n, int) else n)


def _shipped(c, rate):
    return rate * (c + 1) // 4 - rate * c // 4


def _first_bit(c, rate):
    return rate * c % 4 * 8


def _sign_mantissa(a, b):
    low = (a & _i32(0x007F007F)) | (_shr(a, 8) & _i32(0x00800080))
    high = (_shl(b, 8) & _i32(0x7F007F00)) | (b & _i32(0x80008000))
    return low | high


def _exponents(a, b):
    return (_shr(a, 7) & _i32(0x00FF00FF)) | (_shl(b, 1) & _i32(0xFF00FF00))


def _join(sm, e):
    a = (sm & _i32(0x007F007F)) | (_shl(sm, 8) & _i32(0x80008000))
    b = (_shr(sm, 8) & _i32(0x007F007F)) | (sm & _i32(0x80008000))
    return a | (_shl(e, 7) & _i32(0x7F807F80)), b | (_shr(e, 1) & _i32(0x7F807F80))


def _rank(d):
    ge16 = _shr(d + _bytes(128 - 16), 5) & _bytes(4)
    d = ((d + _bytes(12) + ge16) & _bytes(15)) | (d & _bytes(48))
    ge1 = _shr(d + _bytes(128 - 1), 7) & _bytes(1)
    ge5 = _shr(d + _bytes(128 - 5), 7) & _bytes(1)
    return d + _bytes(4) + ge5 - (_shl(ge1, 2) + ge1)


def _unrank(r):
    ge4 = (r + _bytes(128 - 4)) & _bytes(128)
    ge5 = (r + _bytes(128 - 5)) & _bytes(128)
    d = r + _bytes(1) + _shr(ge5, 5) - (_shr(ge4, 5) + _shr(ge4, 7))
    lt16 = _shr(_bytes(128 + 15) - d, 5) & _bytes(4)
    return ((d + lt16) & _bytes(15)) | (d & _bytes(48))


def _encode(exps, base):
    plain = seen = None
    unary = []
    for i, e in enumerate(exps):
        d = base - e
        seen = d if seen is None else seen | d
        r = _rank(d)
        bit = _shl(r & _bytes(1), i) if i else r & _bytes(1)
        plain = bit if plain is None else plain | bit
        unary.append(_shr(r, 1) & _bytes(31))

    strings = []
    longest = None
    for group in (unary[:4], unary[4:]):
        lo = hi = total = None
        for z in reversed(group):
            n = z + _shr(z, 16)
            n = ((n + _shr(n, 8)) & 0xFF) + 4
            longest = n if longest is None else jnp.maximum(longest, n)
            total = n if total is None else total + n
            if lo is not None:
                spilled = _shr(lo, (32 - n) & 31)
                hi = spilled if hi is None else _shl(hi, n & 31) | spilled
            for k in reversed(range(4)):
                lo = jnp.ones_like(z) if lo is None else _shl(lo, 1) | 1
                lo = _shl(lo, (_shr(z, 8 * k) if k else z) & 31)
        longest = jnp.maximum(longest, _shr(total, 1))
        strings.append((lo, hi, total))
    return plain, strings, (seen & _bytes(0xC0)) | _shr(longest, 5)


def _append(strings, waiting, end, c, rate):
    stream = list(waiting) + [None] * SHIPPED
    behind = None
    for g in range(GROUPS):
        lo, hi, total = (v[:, g // 2 * LANES : (g // 2 + 1) * LANES] for v in strings[g % 2])
        first = MIN_RATE * g // 32
        start = jnp.maximum(end, _first_bit(c, rate) + rate * g)
        end = start + total
        skip = _shr(start, 5) - first
        behind = skip if behind is None else behind | skip
        s = start & 31
        back = s ^ 31
        parts = [_shl(lo, s), _shr(_shr(lo, 1), back) | _shl(hi, s), _shr(_shr(hi, 1), back)]
        for d in (1, 2, 4):
            move = (skip & d) != 0
            parts = [
                jnp.where(move, parts[i - d] if i >= d else 0, parts[i] if i < len(parts) else 0)
                for i in range(len(parts) + d)
            ]
        for i, p in enumerate(parts, first):
            stream[i] = p if stream[i] is None else stream[i] | p
    return stream, end, _shr(behind, 3)


def _decode(plain, stream, base, end, c, rate):
    unary = [[None] * GROUPS for _ in range(4)]
    for g in range(GROUPS):
        first = MIN_RATE * g // 32
        start = jnp.maximum(end, _first_bit(c, rate) + rate * g)
        skip = _shr(start, 5) - first
        parts = stream[first:]
        for d in (4, 2, 1):
            move = (skip & d) != 0
            parts = [jnp.where(move, parts[i + d], parts[i]) for i in range(d + 2)]
        s = start & 31
        back = s ^ 31
        lo = _shr(parts[0], s) | _shl(_shl(parts[1], 1), back)
        hi = _shr(parts[1], s) | _shl(_shl(parts[2], 1), back)
        end = start
        for q in range(4):
            rest, ones = lo, None
            for k in range(4):
                cleared = rest & (rest - 1)
                one = pltpu.bitcast((rest ^ cleared).astype(jnp.float32), jnp.int32)
                one = _shr(one, 23 - 8 * k) if k < 3 else _shl(one, 1)
                rest, ones = cleared, one if ones is None else ones | one
            unary[q][g] = ones - _shl(ones, 8) - _i32(0x0101017F)
            n = _shr(ones, 24) - 126
            end = end + n
            if q < 3:
                lo = _shr(lo, n) | _shl(hi, 32 - n)
            if q < 2:
                hi = _shr(hi, n)
    exps = []
    for i in range(8):
        z = jnp.concatenate(unary[i % 4][i // 4 :: 2], axis=1)
        bit = (_shr(plain, i) if i else plain) & _bytes(1)
        exps.append(base - _unrank(_shl(z, 1) | bit))
    return exps, end


PIECE = 128
FAR, NEAR = 9, 7
LOADS, SENDS, RECVS = 3, 2, 4

PLAIN, SIGNS, TAIL, LAST, VERBATIM, END = 8, 12, 24, 34, 44, 76

SENT, KEPT, FROM_Y, FROM_X = range(4)


def _kernel(
    x_ref, far_ref, near_ref,
    in_buf, send_buf, y_buf, x_buf, waiting_ref, end_ref, base_ref, rate_ref, verbatim_ref,
    in_sem, out_sem, y_send, y_recv, x_send, x_recv, y_free, x_free,
):
    shard, n = x_ref.shape
    pieces = shard // 2 // PIECE
    chunks = pieces // 2
    segments = pieces // (FAR + NEAR)
    far_chunks = segments * FAR // 2
    wide = n // LANES

    my_x, my_y = lax.axis_index("x"), lax.axis_index("y")
    y_peer = dict(device_id=(my_x, 1 - my_y), device_id_type=pl.DeviceIdType.MESH)
    x_peer = dict(device_id=(1 - my_x, my_y), device_id_type=pl.DeviceIdType.MESH)
    half = (my_x, 1 - my_x, my_x, 1 - my_x)
    quarter = [2 * y + h for y, h in zip((my_y, my_y, 1 - my_y, 1 - my_y), half)]

    def rows(i):
        return pl.ds(pl.multiple_of(i * PIECE, PIECE), PIECE)

    def blocks(first, count=1):
        return pl.ds(first * LANES, count * LANES)

    def zeros(count=1):
        return jnp.zeros((8, count * LANES), jnp.int32)

    def split(v, count):
        return [v[:, i : i + count * LANES] for i in range(0, v.shape[1], count * LANES)]

    def side_by_side(values):
        return jnp.concatenate(values, axis=1)

    def anywhere(mask):
        return jnp.max(jnp.where(mask, 1, 0))

    def when_chunk(c):
        return pl.when((c >= 0) & (c < chunks))


    def load(s, c, i):
        u = 2 * c + i
        v = jnp.maximum(u - 2 * far_chunks, 0)
        piece = jnp.where(
            c < far_chunks,
            u // FAR * (FAR + NEAR) + u % FAR,
            v // NEAR * (FAR + NEAR) + FAR + v % NEAR,
        )
        return pltpu.make_async_copy(
            x_ref.at[rows(half[s] * pieces + piece)],
            in_buf.at[s, c % LOADS, rows(i)],
            in_sem.at[s, c % LOADS, i],
        )

    def prefetch(s, c):
        @pl.when(c + LOADS < chunks)
        def _():
            for i in range(2):
                load(s, c + LOADS, i).start()

    def result(s, c, i):
        v = 2 * (jnp.where(c < far_chunks, chunks - 2 + c % 2, c) - far_chunks) + i
        return near_ref.at[quarter[s] * segments + v // NEAR, rows(v % NEAR)]

    def store(s, c, i):
        u = 2 * c + i
        return pltpu.make_async_copy(
            result(s, c, i),
            far_ref.at[quarter[s] * segments + u // FAR, rows(u % FAR)],
            out_sem.at[s, c % 2, i],
        )

    def before_result(s, c):
        @pl.when((c >= 2) & (c < far_chunks + 2))
        def _():
            for i in range(2):
                store(s, c - 2, i).wait()

    def after_result(s, c):
        @pl.when(c < far_chunks)
        def _():
            for i in range(2):
                store(s, c, i).start()

    def rounded(s, c, i):
        return in_buf[s, c % LOADS, rows(i)].astype(jnp.bfloat16)


    def to_y(c, lo, hi, part=0):
        return pltpu.make_async_remote_copy(
            send_buf.at[c % SENDS, :, blocks(lo, hi - lo)],
            y_buf.at[c % RECVS, :, blocks(lo, hi - lo)],
            y_send.at[int(lo >= VERBATIM), c % SENDS],
            y_recv.at[part, c % RECVS],
            **y_peer,
        )

    def to_x(c, lo, hi):
        return pltpu.make_async_remote_copy(
            y_buf.at[c % RECVS, :, blocks(lo, hi - lo)],
            x_buf.at[c % RECVS, :, blocks(lo, hi - lo)],
            x_send.at[int(lo >= VERBATIM), c % RECVS],
            x_recv.at[int(lo >= TAIL) + int(lo >= VERBATIM), c % RECVS],
            **x_peer,
        )

    def from_start(s, c, fn):
        start = jnp.where(c == 0, 0, SHIPPED - _shipped(c, rate_ref[s]))
        for lo in range(3):
            pl.when(start == lo)(lambda: fn(lo))

    def by_shipped(count, choices):
        fewer = jnp.where(count == SHIPPED - 1, choices[1], choices[2])
        return jnp.where(count == SHIPPED, choices[0], fewer)

    def begin(s, base):
        end_ref[s] = zeros() + 16
        base = base | _shl(base, 8)
        base_ref[s] = base | _shl(base, 16)

    def read_head(s, buf, c):
        slot = c % RECVS

        @pl.when(c == 0)
        def _():
            head = buf[0, :, blocks(SHIPPED - 1)]
            begin(s, side_by_side([head & 0xFF] * wide))
            rate_ref[s] = jnp.max(_shr(head, 8) & 0xFF)

        first = by_shipped(_shipped(c, rate_ref[s]), split(buf[slot, :, blocks(0, 3)], 1))
        verbatim_ref[s, slot] = anywhere(first == 0)


    def pack(c):
        slot = c % SENDS

        def pairs_of(piece):
            words = pltpu.bitcast(piece, jnp.int32)
            return [(words[i : i + 8], words[i + 8 : i + 16]) for i in range(0, PIECE // 2, 16)]

        @pl.when(c >= SENDS)
        def _():
            sent = c - SENDS
            from_start(SENT, sent, lambda lo: to_y(sent, lo, VERBATIM).wait_send())
            pl.when(verbatim_ref[SENT, slot] != 0)(lambda: to_y(sent, VERBATIM, END).wait_send())

        @when_chunk(c)
        def _():
            early = (TAIL - SIGNS) // wide
            load(SENT, c, 0).wait()
            send_buf[slot, :, blocks(SIGNS, TAIL - SIGNS)] = side_by_side(
                [_sign_mantissa(*p) for p in pairs_of(rounded(SENT, c, 0))[:early]]
            )
            pl.when(c == 0)(lambda: pl.semaphore_wait(barrier, 2))
            pl.when(c >= RECVS)(lambda: pl.semaphore_wait(y_free.at[c % RECVS], 1))
            to_y(c, SIGNS, TAIL, 0).start()

            @pl.when(c == 0)
            def _():
                e = _exponents(*pairs_of(rounded(SENT, c, 0))[0])
                total = jnp.sum((e & 0xFF) + _shr(e, 24))
                mean = (total + 15 * n) // (16 * n)
                begin(SENT, jnp.full_like(e, jnp.clip(mean + 6, 64, 255)))

            load(SENT, c, 1).wait()
            before_result(SENT, c)
            pairs = []
            for i in range(2):
                piece = rounded(SENT, c, i)
                result(SENT, c, i)[...] = piece
                pairs += pairs_of(piece)
            send_buf[slot, :, blocks(TAIL, VERBATIM - TAIL)] = side_by_side(
                [_sign_mantissa(*p) for p in pairs[early:]]
            )
            plain, strings, misfit = _encode([_exponents(*p) for p in pairs], base_ref[SENT])
            send_buf[slot, :, blocks(PLAIN, wide)] = plain

            total = jnp.sum(strings[0][2] + strings[1][2])
            fitting = jnp.clip((total + 26 * n - 1) // (16 * n), MIN_RATE, MAX_RATE)
            rate = jnp.where(c == 0, fitting, rate_ref[SENT])
            rate_ref[SENT] = rate
            waiting = split(waiting_ref[...], 1)
            head = (base_ref[SENT, :, blocks(0)] & 0xFF) | (rate * 256)
            waiting[0] = jnp.where(c == 0, head, waiting[0])

            stream, end, bad = _append(strings, waiting, end_ref[SENT], c, rate)
            count = _shipped(c, rate)
            send_buf[slot, :, blocks(0, SHIPPED)] = side_by_side(stream[:SHIPPED][::-1])
            waiting_ref[...] = by_shipped(
                count, [side_by_side(stream[SHIPPED - k :][:WAITING]) for k in range(3)]
            )
            end = jnp.maximum(end - 32 * count, 0)
            end_ref[SENT] = end
            room = 32 * (_shipped(c + 1, rate) - 1)
            first = by_shipped(count, [stream[SHIPPED - 1 - k] for k in range(3)])
            for block in split(misfit, 1):
                bad = bad | block
            verbatim = anywhere((bad != 0) | (end > room) | (first == 0))
            verbatim_ref[SENT, slot] = verbatim

            @pl.when(verbatim != 0)
            def _():
                send_buf[slot, :, blocks(0, SHIPPED)] = side_by_side([zeros()] + waiting[::-1])
                waiting_ref[...] = zeros(WAITING)
                end_ref[SENT] = zeros()
                send_buf[slot, :, blocks(VERBATIM, END - VERBATIM)] = side_by_side(
                    [_exponents(*p) for i in range(2) for p in pairs_of(rounded(SENT, c, i))]
                )

            from_start(SENT, c, lambda lo: to_y(c, lo, SIGNS, 1).start())
            to_y(c, TAIL, LAST, 2).start()
            to_y(c, LAST, VERBATIM, 3).start()
            pl.when(verbatim != 0)(lambda: to_y(c, VERBATIM, END, 4).start())
            after_result(SENT, c)
            prefetch(SENT, c)

        @pl.when(c == chunks)
        def _():
            send_buf[slot, :, blocks(1, WAITING)] = side_by_side(split(waiting_ref[...], 1)[::-1])
            pl.semaphore_wait(y_free.at[c % RECVS], 1)
            from_start(SENT, c, lambda lo: to_y(c, lo + 1, PLAIN, 1).start())

    def keep(c):
        @when_chunk(c)
        def _():
            for i in range(2):
                load(KEPT, c, i).wait()
            before_result(KEPT, c)
            for i in range(2):
                result(KEPT, c, i)[...] = rounded(KEPT, c, i)
            after_result(KEPT, c)
            prefetch(KEPT, c)

    def pass_on(c, part):
        def one(lo, hi, part):
            to_y(c, lo, hi, part).wait_recv()
            to_x(c, lo, hi).start()

        @when_chunk(c)
        def _():
            if part == 0:
                pl.when(c >= RECVS)(lambda: pl.semaphore_wait(x_free.at[c % RECVS], 1))
                one(SIGNS, TAIL, 0)
            elif part == 1:
                from_start(FROM_Y, c, lambda lo: one(lo, SIGNS, 1))
                read_head(FROM_Y, y_buf, c)
            elif part == 2:
                one(TAIL, LAST, 2)
            else:
                one(LAST, VERBATIM, 3)
                pl.when(verbatim_ref[FROM_Y, c % RECVS] != 0)(lambda: one(VERBATIM, END, 4))

        if part == 1:

            @pl.when(c == chunks)
            def _():
                pl.semaphore_wait(x_free.at[c % RECVS], 1)
                from_start(FROM_Y, c, lambda lo: one(lo + 1, PLAIN, 1))

    def unpack(s, buf, c):
        slot = c % RECVS

        def finish(exps):
            signs = split(buf[slot, :, blocks(SIGNS, VERBATIM - SIGNS)], wide)
            words = [word for sm, e in zip(signs, exps) for word in _join(sm, e)]
            for i in range(2):
                piece = jnp.concatenate(words[8 * i : 8 * i + 8], axis=0)
                result(s, c, i)[...] = pltpu.bitcast(piece, jnp.bfloat16)

        before_result(s, c)
        verbatim = verbatim_ref[s, slot]

        @pl.when(verbatim == 0)
        def _():
            rate = rate_ref[s]
            count = _shipped(c, rate)
            mine = split(buf[slot, :, blocks(0, SHIPPED)], 1)[::-1]
            later = split(buf[(c + 1) % RECVS, :, blocks(1, WAITING)], 1)[::-1]
            joined = [mine[: SHIPPED - k] + later + later[:k] for k in range(3)]
            stream = mine[: SHIPPED - 2] + [
                by_shipped(count, choices) for choices in list(zip(*joined))[SHIPPED - 2 :]
            ]
            plain = buf[slot, :, blocks(PLAIN, wide)]
            exps, end = _decode(plain, stream, base_ref[s], end_ref[s], c, rate)
            end_ref[s] = jnp.maximum(end - 32 * count, 0)
            finish(exps)

        @pl.when(verbatim != 0)
        def _():
            end_ref[s] = zeros()
            finish(split(buf[slot, :, blocks(VERBATIM, END - VERBATIM)], wide))

        after_result(s, c)

    def receive_y(c):
        when_chunk(c)(lambda: unpack(FROM_Y, y_buf, c))

    def free_y(c):
        @when_chunk(c)
        def _():
            slot = c % RECVS
            from_start(FROM_Y, c, lambda lo: to_x(c, lo, VERBATIM).wait_send())
            pl.when(verbatim_ref[FROM_Y, slot] != 0)(lambda: to_x(c, VERBATIM, END).wait_send())
            pl.when(c + RECVS <= chunks)(lambda: pl.semaphore_signal(y_free.at[slot], 1, **y_peer))

    def receive_x(c):
        @when_chunk(c)
        def _():
            to_x(c, TAIL, VERBATIM).wait_recv()
            verbatim = verbatim_ref[FROM_X, c % RECVS]
            pl.when(verbatim != 0)(lambda: to_x(c, VERBATIM, END).wait_recv())

        @when_chunk(c + 1)
        def _():
            from_start(FROM_X, c + 1, lambda lo: to_x(c + 1, lo, TAIL).wait_recv())
            read_head(FROM_X, x_buf, c + 1)

        @pl.when(c + 1 == chunks)
        def _():
            from_start(FROM_X, c + 1, lambda lo: to_x(c + 1, lo + 1, PLAIN).wait_recv())

        @when_chunk(c)
        def _():
            slot = c % RECVS
            unpack(FROM_X, x_buf, c)
            pl.when(c + RECVS <= chunks)(lambda: pl.semaphore_signal(x_free.at[slot], 1, **x_peer))


    for c in range(LOADS + 1):
        for s, k in ((SENT, c), (KEPT, c - 1)):
            if 0 <= k < LOADS:
                for i in range(2):
                    load(s, k, i).start()
    for s in range(4):
        rate_ref[s] = MIN_RATE
    waiting_ref[...] = zeros(WAITING)
    for buf in (y_buf, x_buf):
        for slot in range(RECVS):
            buf[slot, :, blocks(0, 2)] = zeros(2)
    barrier = pltpu.get_barrier_semaphore()
    pl.semaphore_signal(barrier, 1, **y_peer)
    pl.semaphore_signal(barrier, 1, **x_peer)

    def step(t, _):
        pass_on(t - 1, 0)
        pack(t)
        pass_on(t - 1, 1)
        receive_y(t - 2)
        pass_on(t - 1, 2)
        free_y(t - 2)
        keep(t - 1)
        pass_on(t - 1, 3)
        receive_x(t - 2)

    lax.fori_loop(0, chunks + 2, step, None)
    from_start(SENT, chunks, lambda lo: to_y(chunks, lo + 1, PLAIN).wait_send())
    from_start(FROM_Y, chunks, lambda lo: to_x(chunks, lo + 1, PLAIN).wait_send())


def pallas_dist_ag_xy_y_m65536_n1024_kernel(x: jax.Array):
    shard, n = x.shape
    segments = 2 * shard // (PIECE * (FAR + NEAR))
    dma, regular = pltpu.SemaphoreType.DMA, pltpu.SemaphoreType.REGULAR
    far, near = pl.pallas_call(
        _kernel,
        out_shape=[
            jax.ShapeDtypeStruct((segments, FAR * PIECE, n), jnp.bfloat16),
            pltpu.VMEM((segments, NEAR * PIECE, n), jnp.bfloat16),
        ],
        in_specs=[pl.BlockSpec(memory_space=pl.ANY)],
        out_specs=[pl.BlockSpec(memory_space=pl.ANY), pl.BlockSpec(memory_space=pltpu.VMEM)],
        scratch_shapes=[
            pltpu.VMEM((2, LOADS, 2 * PIECE, n), x.dtype),
            pltpu.VMEM((SENDS, 8, END * LANES), jnp.int32),
            pltpu.VMEM((RECVS, 8, END * LANES), jnp.int32),
            pltpu.VMEM((RECVS, 8, END * LANES), jnp.int32),
            pltpu.VMEM((8, WAITING * LANES), jnp.int32),
            pltpu.VMEM((4, 8, LANES), jnp.int32),
            pltpu.VMEM((4, 8, n), jnp.int32),
            pltpu.SMEM((4,), jnp.int32),
            pltpu.SMEM((4, RECVS), jnp.int32),
            dma((2, LOADS, 2)),
            dma((4, 2, 2)),
            dma((2, SENDS)),
            dma((5, RECVS)),
            dma((2, RECVS)),
            dma((3, RECVS)),
            regular((RECVS,)),
            regular((RECVS,)),
        ],
        compiler_params=pltpu.CompilerParams(collective_id=0),
    )(x)

    def tiles(a):
        a = a.reshape(segments, -1, 8, n // 128, 128).transpose(0, 1, 3, 2, 4)
        return a.reshape(segments, -1, 8, 128)

    out = jnp.concatenate([tiles(far), tiles(near)], axis=1)
    return out.reshape(-1, n // 128, 8, 128).transpose(0, 2, 1, 3).reshape(2 * shard, n)
```
